```python
import numpy as np
kernel_name = 'dist_attn_self_mha_htp_b2_sq128_skv128_d512_hq8_dh64'

def setup_inputs():
    x = np.random.randn(2, 128, 512).astype(np.float32)
    Wq = np.random.randn(512, 2048).astype(np.float32) * 0.02
    Wk = np.random.randn(512, 2048).astype(np.float32) * 0.02
    Wv = np.random.randn(512, 2048).astype(np.float32) * 0.02
    Wo = np.random.randn(2048, 512).astype(np.float32) * 0.02
    return {'x': x, 'Wq': Wq, 'Wk': Wk, 'Wv': Wv, 'Wo': Wo}

def reference(x, Wq, Wk, Wv, Wo):
    B, Sq, Hq, Hkv, Dh = (2, 128, 32, 32, 64)
    Q = (x @ Wq).reshape(B, Sq, Hq, Dh)
    K = (x @ Wk).reshape(B, Sq, Hkv, Dh)
    V = (x @ Wv).reshape(B, Sq, Hkv, Dh)
    Skv = K.shape[1]
    out = np.zeros((B, Sq, Hq, Dh), dtype=np.float32)
    m = np.full((B, Hq, Sq, 1), -np.inf, dtype=np.float32)
    l = np.zeros((B, Hq, Sq, 1), dtype=np.float32)
    for j0 in range(0, Skv, 128):
        Kj = K[:, j0:j0 + 128].copy()
        Vj = V[:, j0:j0 + 128].copy()
        sj = np.einsum('bihd,bjhd->bhij', Q, Kj).astype(np.float32) * 0.125
        mj = sj.max(axis=-1, keepdims=True)
        m_new = np.maximum(m, mj)
        alpha = np.exp(m - m_new)
        pj = np.exp(sj - m_new)
        l = l * alpha + pj.sum(axis=-1, keepdims=True)
        out = out * alpha.transpose(0, 2, 1, 3) + np.einsum('bhij,bjhd->bihd', pj, Vj)
        m = m_new
    out = (out / l.transpose(0, 2, 1, 3)).reshape(B, Sq, Hq * Dh)
    return out @ Wo
```

```python
import contextlib
import jax
import jax.numpy as jnp
from jax import lax
from jax.experimental import pallas as pl
from jax.experimental.pallas import tpu as pltpu

B, S, D = 2, 128, 512
M = B * S
NG = 4
NC = 4
CW = D // NC
QR = 64
BF = jnp.bfloat16
F32 = jnp.float32
U32 = jnp.uint32
MESH = pl.DeviceIdType.MESH
QSCALE = 0.125 * 1.4426950408889634

LOADS_B = [("k", 0, 2, 0, 4), ("k", 2, 4, 0, 4), ("q", 0, 2, 0, 4), ("q", 2, 4, 0, 4), ("v", 0, 2, 0, 4), ("v", 2, 4, 0, 4),
           ("o", 0, 4, 1, 2), ("o", 0, 4, 0, 1), ("o", 0, 4, 3, 1)]
PLAN_B = """W1 k0.02 k1.02 k2.02 k3.02
 | W2 k0.24 k1.24 k2.24 k3.24
 | W3 q0.02 q1.02 q2.02 q3.02
 | W4 q30.24 q00.24 q10.24 q20.24 s30x s00x q01.24 q11.24 s10x s20x q21.24 q31.24
 | W5 s01x s11x s21x s31x v0.02 v1.02 v2.02 v3.02
 | W6 v00.24 v10.24 v20.24 v30.24 v01.24 v11.24 v21.24 v31.24 p00 p10 p20 p30 B
 | W7 o10x~ o20~ G p01~ p11~ p21~ p31~ F
 | W8 o00~ o11~ o21~ o01~ F
 | W9 o30~ o31~ F"""


def make(scopes=False, loads=LOADS_B, plan=PLAN_B, newton=True, summode="mmmxmmmx", n2order="01425367", wsmode=1,
         s3=((0, 1), (0, 2), (1, 1), (1, 2)), s2=((0, 0), (1, 0), (0, 3), (1, 3)), nsub=4):
    def sc(name):
        on = scopes is True or (isinstance(scopes, (tuple, list)) and any(name.startswith(p) for p in scopes))
        return jax.named_scope(name) if on else contextlib.nullcontext()

    SR = QR // nsub
    sm = lambda b, g: summode[b] if len(summode) == 2 else summode[b * NG + g]

    def kernel(x, Wq, Wk, Wv, Wo):
        nl = len(loads)

        def body(x_hbm, wq_hbm, wk_hbm, wv_hbm, wo_hbm, out_ref, *scr):
            wbufs = scr[:nl]
            (x_v, acc, xb, qb, kb, vb, pb, lb, ob, own_f,
             s1, r1, s2b, r2, s3b, r3, lsem, ssem, rsem) = scr[nl:]
            hbm = dict(q=wq_hbm, k=wk_hbm, v=wv_hbm, o=wo_hbm)
            ld = [pltpu.make_async_copy(x_hbm, x_v, lsem.at[0])]
            for i, (w, r0, r1_, g0, n) in enumerate(loads):
                ld.append(pltpu.make_async_copy(hbm[w].at[r0 * 128:r1_ * 128, g0 * 128:(g0 + n) * 128], wbufs[i], lsem.at[i + 1]))
            for c in ld:
                c.start()

            def wt(w, g, k0, k1):
                for i, (w_, r0, r1_, g0, n) in enumerate(loads):
                    if w_ == w and r0 <= k0 and k1 <= r1_ and g0 <= g < g0 + n:
                        return wbufs[i][(k0 - r0) * 128:(k1 - r0) * 128, (g - g0) * 128:(g - g0 + 1) * 128].astype(BF)
                raise ValueError((w, g, k0, k1))

            me = lax.axis_index("i")
            pa = me ^ 1
            pb_ = 3 - me
            dside = [jnp.where((me == 0) | (me == 3), 0, 1), me // 2]
            p1_g = [pa, pb_]
            is_r = me == 0
            is_d = me == 2
            hE = jnp.where(me == 3, 1, 0)
            hL = 1 - hE

            bs = pltpu.get_barrier_semaphore()
            for p in (pa, pb_):
                pl.semaphore_signal(bs, inc=1, device_id=(p,), device_id_type=MESH)

            def lo(r):
                return lax.broadcasted_iota(jnp.int32, (r, 128), 1) < 64

            def rows(b):
                return slice(0, M // 2) if b is None else slice(b * S // 2, (b + 1) * S // 2)

            def rowsf(b):
                return slice(0, M) if b is None else slice(b * S, (b + 1) * S)

            def ldb(ref, *idx):
                return pltpu.bitcast(ref[idx], BF)

            def pk(v):
                return pltpu.bitcast(v.astype(BF), U32)

            def gs(g, n=1):
                return slice(g * 128, (g + n) * 128)

            pending = []
            state = {"defer": False}

            def emit(f):
                if state["defer"]:
                    pending.append(f)
                else:
                    f()

            def proj(w, dst, g, b, k0, k1, scale=None):
                r = jnp.dot(ldb(xb, rows(b), gs(k0, k1 - k0)), wt(w, g, k0, k1), preferred_element_type=F32)
                if k0 > 0:
                    r = r + acc[rowsf(b), gs(g)]
                if k1 < 4:
                    def fin():
                        acc[rowsf(b), gs(g)] = r
                else:
                    if scale is not None:
                        r = r * scale
                    r = pk(r)
                    def fin():
                        dst[rows(b), gs(g)] = r
                emit(fin)

            def scores(g, b, nt):
                R = S // nt
                k = ldb(kb, rows(b), gs(g))
                for t in range(nt):
                    r0 = b * S // 2 + t * R // 2
                    q = qb[r0:r0 + R // 2, gs(g)]
                    z = jnp.zeros_like(q)
                    ls = []
                    for h in range(2):
                        qh = jnp.where(lo(R // 2), q, z) if h == 0 else jnp.where(lo(R // 2), z, q)
                        s = lax.dot_general(pltpu.bitcast(qh, BF), k, (((1,), (1,)), ((), ())),
                                            preferred_element_type=F32)
                        m = jnp.max(s, axis=-1, keepdims=True)
                        p = jnp.exp2(s - m)
                        if sm(b, g) == "x":
                            ls.append(jnp.sum(p, axis=-1, keepdims=True))
                        pb[b * NG + g, h, t * R // 2:(t + 1) * R // 2] = pk(p)
                    if sm(b, g) != "x":
                        continue
                    l2 = jnp.where(lo(R), ls[0], ls[1])
                    r = pl.reciprocal(l2, approx=True)
                    if newton:
                        r = r * (2.0 - l2 * r)
                    lb[b * NG + g, t * R:(t + 1) * R] = r

            def pv(g, b, nt):
                R = S // nt
                if sm(b, g) == "x":
                    v = [ldb(vb, rows(b), gs(g))] * 2
                else:
                    vu = vb[rows(b), gs(g)]
                    one = jnp.full(vu.shape, 0x3F803F80, U32)
                    v = [pltpu.bitcast(jnp.where(lo(S // 2), vu, one), BF), pltpu.bitcast(jnp.where(lo(S // 2), one, vu), BF)]
                for t in range(nt):
                    o2 = [jnp.dot(ldb(pb, b * NG + g, h, slice(t * R // 2, (t + 1) * R // 2)), v[h],
                                  preferred_element_type=F32) for h in range(2)]
                    if sm(b, g) == "x":
                        r = lb[b * NG + g, t * R:(t + 1) * R]
                    else:
                        l2 = pltpu.roll(jnp.where(lo(R), o2[1], o2[0]), 64, 1)
                        r = pl.reciprocal(l2, approx=True)
                        if newton:
                            r = r * (2.0 - l2 * r)
                    o = jnp.where(lo(R), o2[0], o2[1]) * r
                    r0 = b * S // 2 + t * R // 2
                    def fin(o=pk(o), r0=r0):
                        ob[r0:r0 + R // 2, gs(g)] = o
                    emit(fin)

            def rc(ph, sbuf, rbuf, it, j, dev):
                u = it * nsub + j
                idx = ph * 16 * nsub + u
                return pltpu.make_async_remote_copy(
                    src_ref=sbuf.at[u], dst_ref=rbuf.at[u],
                    send_sem=ssem.at[idx], recv_sem=rsem.at[idx],
                    device_id=(dev,), device_id_type=MESH)

            def oproj(c, b, fine):
                own_side = 0 if (b, c) in s3 else 1
                it0 = (b * NC + c) * 2
                if fine:
                    order = [(h, j) for j in range(nsub) for h in range(2)]
                    lhs = jnp.concatenate([ob[pl.ds(b * S // 2 + (h * QR + j * SR) // 2, SR // 2), :] for (h, j) in order], axis=0)
                    pr = jnp.dot(pltpu.bitcast(lhs, BF), wt("o", c, 0, 4), preferred_element_type=F32)
                    part = {hj: pr[n * SR:(n + 1) * SR] for n, hj in enumerate(order)}
                    def finj(j):
                        for h in range(2):
                            s1[(it0 + h) * nsub + j] = part[h, j].astype(BF)
                        for h in range(2):
                            @pl.when(dside[h] != own_side)
                            def _():
                                rc(0, s1, r1, it0 + h, j, p1_g[h]).start()
                    for j in range(nsub):
                        emit(lambda j=j: finj(j))
                    def fin():
                        for (h, j) in order:
                            own_f[(it0 + h) * nsub + j] = part[h, j]
                else:
                    pr = jnp.dot(ldb(ob, rows(b), slice(None)), wt("o", c, 0, 4), preferred_element_type=F32)
                    def fin():
                        for h in range(2):
                            for j in range(nsub):
                                s1[(it0 + h) * nsub + j] = pr[h * QR + j * SR:h * QR + (j + 1) * SR].astype(BF)
                        for j in range(nsub):
                            for h in range(2):
                                @pl.when(dside[h] != own_side)
                                def _():
                                    rc(0, s1, r1, it0 + h, j, p1_g[h]).start()
                        for h in range(2):
                            for j in range(nsub):
                                own_f[(it0 + h) * nsub + j] = pr[h * QR + j * SR:h * QR + (j + 1) * SR]
                emit(fin)

            with sc("a_x"):
                ld[0].wait()
                xb[...] = pk(x_v[...])
            for ri, reg in enumerate(plan.split("|")):
                with sc(f"r{ri + 1:02d}_" + "_".join(reg.replace("~", "d").replace(".", "").split())[:40]):
                    for op in reg.split():
                        state["defer"] = op.endswith("~")
                        op = op.rstrip("~")
                        kind = op[0]
                        if kind == "F":
                            for f in pending:
                                f()
                            pending.clear()
                            continue
                        if kind == "G":
                            pending.pop(0)()
                            continue
                        if kind == "W":
                            with sc(f"r{ri + 1:02d}W"):
                                ld[int(op[1:])].wait()
                            continue
                        if kind == "B":
                            pl.semaphore_wait(bs, 2)
                            continue
                        k0, k1 = 0, 4
                        if "." in op:
                            op, kk = op.split(".")
                            k0, k1 = int(kk[0]), int(kk[1])
                        g = int(op[1])
                        b = int(op[2]) if op[2:3].isdigit() else None
                        one = op.endswith("x")
                        if kind == "q":
                            proj("q", qb, g, b, k0, k1, QSCALE)
                        elif kind == "k":
                            proj("k", kb, g, b, k0, k1)
                        elif kind == "v":
                            proj("v", vb, g, b, k0, k1)
                        elif kind in "sp":
                            f = scores if kind == "s" else pv
                            if b is None:
                                f(g, 0, 1); f(g, 1, 1)
                            else:
                                f(g, b, 1 if one else 2)
                        elif kind == "o":
                            oproj(g, b, one)

            def sel3(r, n, d):
                return jnp.where(is_r, r, jnp.where(is_d, d, n))

            def ch(bc):
                return bc[0] * NC + bc[1]

            def unit(n, r_l, n_l, d_l):
                p, w = n // (2 * nsub), n % (2 * nsub)
                chunk = sel3(ch(r_l[p]), ch(n_l[n][0]), ch(d_l[p]))
                h = sel3(w % 2, n_l[n][1], w % 2)
                j = sel3(w // 2, n_l[n][2], w // 2)
                it = chunk * 2 + h
                p1 = jnp.where(h == 0, pa, pb_)
                p2 = jnp.where(h == 0, pb_, pa)
                row = pl.multiple_of((chunk // NC) * S + h * QR + j * SR, SR)
                col = pl.multiple_of((chunk % NC) * CW, CW)
                return it, j, p1, p2, row, col

            NU = 8 * nsub
            nl2 = []
            for kn in n2order:
                kn = int(kn)
                nl2 += [((s2[kn], hE, j) if kn < 4 else (s3[kn - 4], hL, j)) for j in range(nsub)]
            nl3, nlf = [], []
            for p in range(4):
                nl3 += [(s3[p], hL, j) for j in range(nsub)] + [(s2[p], hE, j) for j in range(nsub)]
                for j in range(nsub):
                    nlf += [(s3[p], hE, j), (s2[p], hL, j)]
            own2 = [unit(n, s3, nl2, s2) for n in range(NU)]
            own3 = [unit(n, s3, nl3, s2) for n in range(NU)]
            oth = [unit(n, s2, nlf, s3) for n in range(NU)]

            sends = []
            for n in range(NU):
                it, j, p1, p2, row, col = own2[n]
                u = it * nsub + j
                with sc(f"g_p2_{n:02d}"):
                    rc(0, s1, r1, it, j, p1).wait_recv()
                    a = own_f[u] + r1[u].astype(F32)
                    s2b[u] = a.astype(BF)
                    d = rc(1, s2b, r2, it, j, p2); d.start(); sends.append(d)
                    own_f[u] = a
            for n in range(NU):
                it, j, p1, p2, row, col = own3[n]
                u = it * nsub + j
                with sc(f"h_p3_{n:02d}"):
                    rc(0, s1, r1, oth[n][0], oth[n][1], oth[n][2]).wait_send()
                    rc(1, s2b, r2, it, j, p2).wait_recv()
                    a = own_f[u] + r2[u].astype(F32)
                    s3b[u] = a.astype(BF)
                    d = rc(2, s3b, r3, it, j, p1); d.start(); sends.append(d)
                    out_ref[pl.ds(row, SR), pl.ds(col, CW)] = a
            for n in range(NU):
                it, j, p1, p2, row, col = oth[n]
                u = it * nsub + j
                with sc(f"i_fin_{n:02d}"):
                    sends[n].wait_send()
                    sends[NU + n].wait_send()
                    rc(2, s3b, r3, it, j, p1).wait_recv()
                    out_ref[pl.ds(row, SR), pl.ds(col, CW)] = r3[u].astype(F32)

        out = pl.pallas_call(
            body,
            out_shape=jax.ShapeDtypeStruct((M, D), F32),
            in_specs=[pl.BlockSpec(memory_space=pl.ANY)] * 5,
            out_specs=pl.BlockSpec(memory_space=pltpu.VMEM),
            scratch_shapes=[pltpu.VMEM((128 * (r1_ - r0), 128 * n), F32) for (_, r0, r1_, _, n) in loads] + [
                pltpu.VMEM((M, D), F32), pltpu.VMEM((M, D), F32),
                pltpu.VMEM((M // 2, D), U32), pltpu.VMEM((M // 2, D), U32), pltpu.VMEM((M // 2, D), U32), pltpu.VMEM((M // 2, D), U32),
                pltpu.VMEM((B * NG, 2, S // 2, 128), U32), pltpu.VMEM((B * NG, S, 128), F32),
                pltpu.VMEM((M // 2, D), U32),
                pltpu.VMEM((16 * nsub, SR, CW), F32),
            ] + [pltpu.VMEM((16 * nsub, SR, CW), BF)] * 6 + [
                pltpu.SemaphoreType.DMA((nl + 1,)),
                pltpu.SemaphoreType.DMA((3 * 16 * nsub,)),
                pltpu.SemaphoreType.DMA((3 * 16 * nsub,)),
            ],
            compiler_params=pltpu.CompilerParams(collective_id=0, disable_semaphore_checks=True, disable_bounds_checks=True),
        )(x.reshape(M, D), Wq, Wk, Wv, Wo)
        return out.reshape(B, S, D)
    return kernel


def pallas_dist_attn_self_mha_htp_b2_sq128_skv128_d512_hq8_dh64_kernel(x, Wq, Wk, Wv, Wo):
    return make()(x, Wq, Wk, Wv, Wo)
```

```python
import jax
import jax.numpy as jnp
from jax import lax
from jax.experimental import pallas as pl
from jax.experimental.pallas import tpu as pltpu

B, S, D = 2, 128, 512
M = B * S
NG = 4
NC = 4
HR = 64
SR = 16
NSUB = HR // SR
NU = B * NC * 2 * NSUB // 2
BF = jnp.bfloat16
F32 = jnp.float32
MESH = pl.DeviceIdType.MESH
QSCALE = 0.125 * 1.4426950408889634

R_SIDE = ((0, 0), (0, 1), (1, 0), (0, 2))
D_SIDE = ((1, 1), (1, 2), (0, 3), (1, 3))


def _dot(a, b):
    return jnp.dot(a, b, preferred_element_type=F32)


def _body(x_hbm, wq_hbm, wk_hbm, wv_hbm, wo_hbm, out_ref,
          x_v, x1_v, wk_v, wq_v, wv_v, wo_v, acc_v, part_v,
          snd1, rcv1, snd2, rcv2, snd3, rcv3,
          ld_sem, x_sem, snd_sem, rcv_sem):
    def wcopy(src, dst, half, s):
        return pltpu.make_async_copy(src.at[pl.ds(half * 256, 256)], dst.at[half], ld_sem.at[s])

    ld_x0 = pltpu.make_async_copy(x_hbm.at[pl.ds(0, S)], x_v.at[pl.ds(0, S)], ld_sem.at[0])
    ld_x1 = [pltpu.make_async_copy(x_hbm.at[pl.ds(S + r * HR, HR)], x_v.at[pl.ds(S + r * HR, HR)],
                                   ld_sem.at[1 + r]) for r in range(2)]
    ld_k = [wcopy(wk_hbm, wk_v, h, 3 + h) for h in range(2)]
    ld_q = [wcopy(wq_hbm, wq_v, h, 5 + h) for h in range(2)]
    ld_v = [wcopy(wv_hbm, wv_v, h, 7 + h) for h in range(2)]
    ld_o = [pltpu.make_async_copy(wo_hbm.at[:, pl.ds(c * 128, 128)], wo_v.at[c], ld_sem.at[9 + c])
            for c in range(NC)]

    ld_x0.start()
    me = lax.axis_index("i")
    is_r = me == 0
    is_d = me == 2
    has_x1 = [is_r | (me == 1), is_r | (me == 3)]
    for r in range(2):
        pl.when(has_x1[r])(ld_x1[r].start)
    ld_k[0].start()

    nbr = [me ^ 1, 3 - me]
    barrier = pltpu.get_barrier_semaphore()
    for p in nbr:
        pl.semaphore_signal(barrier, inc=1, device_id=(p,), device_id_type=MESH)
    for cp in (ld_q[0], ld_k[1], ld_q[1], ld_v[0], ld_v[1], *ld_o):
        cp.start()

    d_side = [jnp.where(is_r | (me == 3), 0, 1), me // 2]
    h_early = jnp.where(me == 3, 1, 0)
    h_late = 1 - h_early

    def unit_list(r_chunks, n_units, d_chunks):
        res = []
        for n in range(NU):
            p, w = divmod(n, 2 * NSUB)
            (nb, nc), nh, nj = n_units[n]

            def pick(r, nn, d):
                return jnp.where(is_r, r, jnp.where(is_d, d, nn))
            b = pick(r_chunks[p][0], nb, d_chunks[p][0])
            c = pick(r_chunks[p][1], nc, d_chunks[p][1])
            h = pick(w % 2, nh, w % 2)
            j = pick(w // 2, nj, w // 2)
            uid = ((b * NC + c) * 2 + h) * NSUB + j
            row = pl.multiple_of(b * S + h * HR + j * SR, SR)
            col = pl.multiple_of(c * 128, 128)
            res.append((uid, h, row, col))
        return res

    n_own, n_fin = [], []
    n_own3 = []
    for p in range(4):
        n_own += [(D_SIDE[p], h_early, j) for j in range(NSUB)] + [(R_SIDE[p], h_late, j) for j in range(NSUB)]
        n_own3 += [(R_SIDE[p], h_late, j) for j in range(NSUB)] + [(D_SIDE[p], h_early, j) for j in range(NSUB)]
        for j in range(NSUB):
            n_fin += [(R_SIDE[p], h_early, j), (D_SIDE[p], h_late, j)]
    own2 = unit_list(R_SIDE, n_own, D_SIDE)
    own3 = unit_list(R_SIDE, n_own3, D_SIDE)
    other = unit_list(D_SIDE, n_fin, R_SIDE)

    def rcopy(phase, uid, h):
        snd, rcv = ((snd1, rcv1), (snd2, rcv2), (snd3, rcv3))[phase]
        if isinstance(h, int):
            dev = nbr[h] if phase != 1 else nbr[1 - h]
        else:
            dev = jnp.where((h == 0) if phase != 1 else (h == 1), nbr[0], nbr[1])
        return pltpu.make_async_remote_copy(
            src_ref=snd.at[uid], dst_ref=rcv.at[uid],
            send_sem=snd_sem.at[phase * 2 * NU + uid], recv_sem=rcv_sem.at[phase * 2 * NU + uid],
            device_id=(dev,), device_id_type=MESH)

    def x1_copy(kh, r):
        return pltpu.make_async_remote_copy(
            src_ref=x1_v.at[kh, r], dst_ref=x1_v.at[kh, r],
            send_sem=x_sem.at[2 + 2 * kh + r], recv_sem=x_sem.at[kh],
            device_id=(jnp.where(is_r, 3 - 2 * r, 2),), device_id_type=MESH)

    def x1_wait(kh):
        @pl.when(is_d)
        def _():
            pltpu.make_async_copy(x1_v.at[kh], x1_v.at[kh], x_sem.at[kh]).wait()

        @pl.when(me % 2 == 1)
        def _():
            x1_copy(kh, 1 - me // 2).wait_recv()
        return jnp.concatenate(
            [jnp.concatenate([x1_v[kh, r, t] for r in range(2)], axis=0) for t in range(2)], axis=1)

    def lanes_lo(rows):
        return lax.broadcasted_iota(jnp.int32, (rows, 128), 1) < 64

    def proj(xh, w, b, half, g):
        res = _dot(xh, (wk_v, wq_v, wv_v)[w][half, :, g * 128:(g + 1) * 128].astype(BF))
        if half == 0:
            acc_v[w, b, g] = res
            return None
        return res + acc_v[w, b, g]

    def probs(q, k):
        res = []
        for h in range(2):
            qh = jnp.where(lanes_lo(S), q, 0.0) if h == 0 else jnp.where(lanes_lo(S), 0.0, q)
            s = lax.dot_general(qh.astype(BF), k, (((1,), (1,)), ((), ())), preferred_element_type=F32)
            res.append(jnp.exp2(s - jnp.max(s, axis=-1, keepdims=True)).astype(BF))
        return res

    def inv_sum(p):
        l = jnp.where(lanes_lo(S), *[jnp.sum(ph.astype(F32), axis=-1, keepdims=True) for ph in p])
        r = pl.reciprocal(l, approx=True)
        return r * (2.0 - l * r)

    def attend(p, v, r, tiles):
        rows = S // tiles
        res = []
        for t in range(tiles):
            sl = slice(t * rows, (t + 1) * rows)
            o = jnp.where(lanes_lo(rows), _dot(p[0][sl], v), _dot(p[1][sl], v))
            res.append((o * r[sl]).astype(BF))
        return res[0] if tiles == 1 else jnp.concatenate(res, axis=0)

    def out_proj(o, b, c):
        order = [(h, j) for j in range(NSUB) for h in range(2)]
        lhs = jnp.concatenate([o[h * HR + j * SR:h * HR + (j + 1) * SR] for h, j in order], axis=0)
        res = _dot(lhs, wo_v[c].astype(BF))
        piece = {hj: res[n * SR:(n + 1) * SR] for n, hj in enumerate(order)}
        uid = {(h, j): ((b * NC + c) * 2 + h) * NSUB + j for h, j in order}
        owner_side = 0 if (b, c) in R_SIDE else 1

        def publish(j):
            for h in range(2):
                snd1[uid[h, j]] = piece[h, j].astype(BF)
            for h in range(2):
                pl.when(d_side[h] != owner_side)(rcopy(0, uid[h, j], h).start)

        def keep():
            for hj in order:
                part_v[uid[hj]] = piece[hj]
        return [lambda j=j: publish(j) for j in range(NSUB)], keep

    G = range(NG)

    ld_x0.wait()
    x0 = [x_v[0:S, kh * 256:(kh + 1) * 256].astype(BF) for kh in range(2)]
    for r in range(2):
        @pl.when(has_x1[r])
        def _():
            ld_x1[r].wait()
            for kh in range(2):
                for t in range(2):
                    c0 = kh * 256 + t * 128
                    x1_v[kh, r, t] = x_v[S + r * HR:S + (r + 1) * HR, c0:c0 + 128].astype(BF)
    pl.semaphore_wait(barrier, 2)
    for kh in range(2):
        for r in range(2):
            pl.when(has_x1[r])(x1_copy(kh, r).start)

    WK, WQ, WV = range(3)
    ld_k[0].wait()
    for g in G:
        proj(x0[0], WK, 0, 0, g)
    ld_q[0].wait()
    for g in G:
        proj(x0[0], WQ, 0, 0, g)
    x1 = [x1_wait(0)]
    for w in (WK, WQ):
        for g in G:
            proj(x1[0], w, 1, 0, g)
    ld_k[1].wait()
    k0 = [proj(x0[1], WK, 0, 1, g).astype(BF) for g in G]
    x1.append(x1_wait(1))
    k1 = [proj(x1[1], WK, 1, 1, g).astype(BF) for g in G]
    ld_q[1].wait()
    q0 = [proj(x0[1], WQ, 0, 1, g) * QSCALE for g in G]
    p0 = [probs(q0[g], k0[g]) for g in G]
    q1 = [proj(x1[1], WQ, 1, 1, g) * QSCALE for g in G]

    ld_v[0].wait()
    r0 = [inv_sum(p0[g]) for g in G]
    for g in (0, 1):
        proj(x0[0], WV, 0, 0, g)
    p1 = [probs(q1[g], k1[g]) for g in G]
    for b, g in ((0, 2), (0, 3), (1, 0), (1, 1), (1, 2), (1, 3)):
        proj((x0, x1)[b][0], WV, b, 0, g)
    ld_v[1].wait()
    r1 = [inv_sum(p1[g]) for g in G]
    v0 = [proj(x0[1], WV, 0, 1, g).astype(BF) for g in G]
    v1 = [proj(x1[1], WV, 1, 1, g).astype(BF) for g in (0, 1)]
    o0 = jnp.concatenate([attend(p0[g], v0[g], r0[g], 1 if g < 2 else 2) for g in G], axis=1)

    ld_o[0].wait()
    pub, keep = out_proj(o0, 0, 0)
    v1 += [proj(x1[1], WV, 1, 1, g).astype(BF) for g in (2, 3)]
    pub[0]()
    o1 = [attend(p1[0], v1[0], r1[0], 2)]
    for f in (*pub[1:], keep):
        f()

    def two_chunks(a, b):
        for f in (*a[0], *b[0], a[1], b[1]):
            f()

    ld_o[1].wait()
    pub, keep = out_proj(o0, 0, 1)
    o1 += [attend(p1[g], v1[g], r1[g], 2) for g in (1, 2)]
    pub[0]()
    o1.append(attend(p1[3], v1[3], r1[3], 2))
    for f in (*pub[1:], keep):
        f()
    o1 = jnp.concatenate(o1, axis=1)
    two_chunks(out_proj(o1, 1, 1), out_proj(o1, 1, 0))
    ld_o[2].wait()
    two_chunks(out_proj(o1, 1, 2), out_proj(o0, 0, 2))
    ld_o[3].wait()
    two_chunks(out_proj(o0, 0, 3), out_proj(o1, 1, 3))

    for kh in range(2):
        for r in range(2):
            pl.when(has_x1[r])(x1_copy(kh, r).wait_send)

    for uid, h, _, _ in own2:
        rcopy(0, uid, h).wait_recv()
        acc = part_v[uid] + rcv1[uid].astype(F32)
        snd2[uid] = acc.astype(BF)
        rcopy(1, uid, h).start()
        part_v[uid] = acc
    for n, (uid, h, row, col) in enumerate(own3):
        rcopy(0, other[n][0], other[n][1]).wait_send()
        rcopy(1, uid, h).wait_recv()
        acc = part_v[uid] + rcv2[uid].astype(F32)
        snd3[uid] = acc.astype(BF)
        rcopy(2, uid, h).start()
        out_ref[pl.ds(row, SR), pl.ds(col, 128)] = acc
    for n, (uid, h, row, col) in enumerate(other):
        rcopy(1, own2[n][0], own2[n][1]).wait_send()
        rcopy(2, own3[n][0], own3[n][1]).wait_send()
        rcopy(2, uid, h).wait_recv()
        out_ref[pl.ds(row, SR), pl.ds(col, 128)] = rcv3[uid].astype(F32)


def pallas_dist_attn_self_mha_htp_b2_sq128_skv128_d512_hq8_dh64_kernel(x, Wq, Wk, Wv, Wo):
    unit_buf = pltpu.VMEM((2 * NU, SR, 128), BF)
    out = pl.pallas_call(
        _body,
        out_shape=jax.ShapeDtypeStruct((M, D), F32),
        in_specs=[pl.BlockSpec(memory_space=pl.ANY)] * 5,
        out_specs=pl.BlockSpec(memory_space=pltpu.VMEM),
        scratch_shapes=[
            pltpu.VMEM((M, D), F32),
            pltpu.VMEM((2, 2, 2, HR, 128), BF),
            pltpu.VMEM((2, 256, D), F32),
            pltpu.VMEM((2, 256, D), F32),
            pltpu.VMEM((2, 256, D), F32),
            pltpu.VMEM((NC, D, 128), F32),
            pltpu.VMEM((3, B, NG, S, 128), F32),
            pltpu.VMEM((2 * NU, SR, 128), F32),
            unit_buf, unit_buf, unit_buf, unit_buf, unit_buf, unit_buf,
            pltpu.SemaphoreType.DMA((9 + NC,)),
            pltpu.SemaphoreType.DMA((6,)),
            pltpu.SemaphoreType.DMA((3 * 2 * NU,)),
            pltpu.SemaphoreType.DMA((3 * 2 * NU,)),
        ],
        compiler_params=pltpu.CompilerParams(
            collective_id=0, disable_semaphore_checks=True, disable_bounds_checks=True),
    )(x.reshape(M, D), Wq, Wk, Wv, Wo)
    return out.reshape(B, S, D)
```

```python
import jax
import jax.numpy as jnp
from jax import lax
from jax.experimental import pallas as pl
from jax.experimental.pallas import tpu as pltpu

B, S, D = 2, 128, 512
M = B * S
NG = 4
NC = 4
HR = 64
SR = 16
NSUB = HR // SR
NU = B * NC * 2 * NSUB
BF = jnp.bfloat16
F32 = jnp.float32
MESH = pl.DeviceIdType.MESH
QSCALE = 0.125 * 1.4426950408889634


def _blocks(b, c, js=range(NSUB)):
    return [(b, c, j) for j in js]


R_SIDE = _blocks(0, 0) + _blocks(0, 1) + _blocks(1, 1, [3]) + _blocks(1, 0) + _blocks(0, 2)
D_SIDE = _blocks(1, 1, [0, 1, 2]) + _blocks(1, 2) + _blocks(0, 3) + _blocks(1, 3)
ROW_ORDER = [(h, j) for j in range(NSUB) for h in range(2)]


def _dot(a, b):
    return jnp.dot(a, b, preferred_element_type=F32)


def _body(x_hbm, wq_hbm, wk_hbm, wv_hbm, wo_hbm, out_ref,
          x_v, x1_v, wk_v, wq_v, wv_v, wo_v, acc_v, part_v,
          snd1, rcv1, snd2, rcv2, snd3, rcv3,
          ld_sem, x_sem, snd_sem, rcv_sem):
    def wcopy(src, dst, half, s):
        return pltpu.make_async_copy(src.at[pl.ds(half * 256, 256)], dst.at[half], ld_sem.at[s])

    ld_x0 = pltpu.make_async_copy(x_hbm.at[pl.ds(0, S)], x_v.at[pl.ds(0, S)], ld_sem.at[0])
    ld_x1 = [pltpu.make_async_copy(x_hbm.at[pl.ds(S + r * HR, HR)], x_v.at[pl.ds(S + r * HR, HR)],
                                   ld_sem.at[1 + r]) for r in range(2)]
    ld_k = [wcopy(wk_hbm, wk_v, h, 3 + h) for h in range(2)]
    ld_q = [wcopy(wq_hbm, wq_v, h, 5 + h) for h in range(2)]
    ld_v = [wcopy(wv_hbm, wv_v, h, 7 + h) for h in range(2)]
    ld_o = [pltpu.make_async_copy(wo_hbm.at[:, pl.ds(c * 128, 128)], wo_v.at[c], ld_sem.at[9 + c])
            for c in range(NC)]

    ld_x0.start()
    me = lax.axis_index("i")
    is_r = me == 0
    is_d = me == 2
    has_x1 = [is_r | (me == 1), is_r | (me == 3)]
    for r in range(2):
        pl.when(has_x1[r])(ld_x1[r].start)
    ld_k[0].start()

    nbr = [me ^ 1, 3 - me]
    barrier = pltpu.get_barrier_semaphore()
    for p in nbr:
        pl.semaphore_signal(barrier, inc=1, device_id=(p,), device_id_type=MESH)
    for cp in (ld_q[0], ld_k[1], ld_q[1], ld_v[0], ld_v[1], *ld_o):
        cp.start()

    d_side = [jnp.where(is_r | (me == 3), 0, 1), me // 2]
    h_early = jnp.where(me == 3, 1, 0)
    h_late = 1 - h_early

    def unit_list(r_blocks, n_units, d_blocks, pad_front=False):
        both = lambda blocks: [(blk, h) for blk in blocks for h in range(2)]
        lists = (both(r_blocks), n_units, both(d_blocks))
        res = []
        total = max(map(len, lists))
        for n in range(total):
            pos = [n - (total - len(l)) if pad_front else n for l in lists]
            ent = [l[min(max(i, 0), len(l) - 1)] for l, i in zip(lists, pos)]

            def pick(f):
                r, nn, d = map(f, ent)
                return jnp.where(is_r, r, jnp.where(is_d, d, nn))
            ok = [0 <= i < len(l) for l, i in zip(lists, pos)]
            valid = None if all(ok) else jnp.where(is_r, ok[0], jnp.where(is_d, ok[2], ok[1]))
            b, c, j = (pick(lambda e, i=i: e[0][i]) for i in range(3))
            h = pick(lambda e: e[1])
            uid = ((b * NC + c) * 2 + h) * NSUB + j
            row = pl.multiple_of(b * S + h * HR + j * SR, SR)
            col = pl.multiple_of(c * 128, 128)
            res.append((valid, uid, h, row, col))
        return res

    def interleave(a, b, k):
        res = []
        for i in range(0, max(len(a), len(b)), k):
            res += a[i:i + k] + b[i:i + k]
        return res

    tag = lambda blocks, h: [(blk, h) for blk in blocks]
    own2 = unit_list(R_SIDE, interleave(tag(D_SIDE, h_early), tag(R_SIDE, h_late), NSUB), D_SIDE)
    own3 = unit_list(R_SIDE, interleave(tag(R_SIDE, h_late), tag(D_SIDE, h_early), NSUB), D_SIDE)
    other = unit_list(D_SIDE, interleave(tag(R_SIDE, h_early), tag(D_SIDE, h_late), 1), R_SIDE, True)

    def when(valid, f):
        if valid is None:
            f()
        else:
            pl.when(valid)(f)

    def rcopy(phase, uid, h):
        snd, rcv = ((snd1, rcv1), (snd2, rcv2), (snd3, rcv3))[phase]
        if isinstance(h, int):
            dev = nbr[h] if phase != 1 else nbr[1 - h]
        else:
            dev = jnp.where((h == 0) if phase != 1 else (h == 1), nbr[0], nbr[1])
        return pltpu.make_async_remote_copy(
            src_ref=snd.at[uid], dst_ref=rcv.at[uid],
            send_sem=snd_sem.at[phase * NU + uid], recv_sem=rcv_sem.at[phase * NU + uid],
            device_id=(dev,), device_id_type=MESH)

    def x1_copy(kh, r):
        return pltpu.make_async_remote_copy(
            src_ref=x1_v.at[kh, r], dst_ref=x1_v.at[kh, r],
            send_sem=x_sem.at[2 + 2 * kh + r], recv_sem=x_sem.at[kh],
            device_id=(jnp.where(is_r, 3 - 2 * r, 2),), device_id_type=MESH)

    def x1_wait(kh):
        @pl.when(is_d)
        def _():
            pltpu.make_async_copy(x1_v.at[kh], x1_v.at[kh], x_sem.at[kh]).wait()

        @pl.when(me % 2 == 1)
        def _():
            x1_copy(kh, 1 - me // 2).wait_recv()
        return jnp.concatenate(
            [jnp.concatenate([x1_v[kh, r, t] for r in range(2)], axis=0) for t in range(2)], axis=1)

    def lanes_lo(rows):
        return lax.broadcasted_iota(jnp.int32, (rows, 128), 1) < 64

    def proj(xh, w, b, half, g):
        res = _dot(xh, (wk_v, wq_v, wv_v)[w][half, :, g * 128:(g + 1) * 128].astype(BF))
        if half == 0:
            acc_v[w, b, g] = res
            return None
        return res + acc_v[w, b, g]

    def probs(q, k):
        res = []
        for h in range(2):
            qh = jnp.where(lanes_lo(S), q, 0.0) if h == 0 else jnp.where(lanes_lo(S), 0.0, q)
            s = lax.dot_general(qh.astype(BF), k, (((1,), (1,)), ((), ())), preferred_element_type=F32)
            res.append(jnp.exp2(s - jnp.max(s, axis=-1, keepdims=True)).astype(BF))
        return res

    def inv_sum(p):
        l = jnp.where(lanes_lo(S), *[jnp.sum(ph.astype(F32), axis=-1, keepdims=True) for ph in p])
        r = pl.reciprocal(l, approx=True)
        return r * (2.0 - l * r)

    def attend(p, v, r, tiles):
        rows = S // tiles
        res = []
        for t in range(tiles):
            sl = slice(t * rows, (t + 1) * rows)
            o = jnp.where(lanes_lo(rows), _dot(p[0][sl], v), _dot(p[1][sl], v))
            res.append((o * r[sl]).astype(BF))
        return res[0] if tiles == 1 else jnp.concatenate(res, axis=0)

    def unit_rows(a, t):
        sel = ROW_ORDER[t * NSUB:(t + 1) * NSUB]
        return jnp.concatenate([a[h * HR + j * SR:h * HR + (j + 1) * SR] for h, j in sel], axis=0)

    def attend_tile(p, v, r, t):
        o = jnp.where(lanes_lo(HR), _dot(unit_rows(p[0], t), v), _dot(unit_rows(p[1], t), v))
        return (o * unit_rows(r, t)).astype(BF)

    def out_proj(o, b, c):
        res = _dot(o, wo_v[c].astype(BF))
        piece = {hj: res[n * SR:(n + 1) * SR] for n, hj in enumerate(ROW_ORDER)}
        uid = {(h, j): ((b * NC + c) * 2 + h) * NSUB + j for h, j in ROW_ORDER}

        def publish(j):
            owner_side = 0 if (b, c, j) in R_SIDE else 1
            for h in range(2):
                snd1[uid[h, j]] = piece[h, j].astype(BF)
            for h in range(2):
                pl.when(d_side[h] != owner_side)(rcopy(0, uid[h, j], h).start)
            for h in range(2):
                part_v[uid[h, j]] = piece[h, j]
        return [lambda j=j: publish(j) for j in range(NSUB)]

    G = range(NG)

    ld_x0.wait()
    x0 = [x_v[0:S, kh * 256:(kh + 1) * 256].astype(BF) for kh in range(2)]
    for r in range(2):
        @pl.when(has_x1[r])
        def _():
            ld_x1[r].wait()
            for kh in range(2):
                for t in range(2):
                    c0 = kh * 256 + t * 128
                    x1_v[kh, r, t] = x_v[S + r * HR:S + (r + 1) * HR, c0:c0 + 128].astype(BF)
    pl.semaphore_wait(barrier, 2)
    for kh in range(2):
        for r in range(2):
            pl.when(has_x1[r])(x1_copy(kh, r).start)

    WK, WQ, WV = range(3)
    ld_k[0].wait()
    for g in G:
        proj(x0[0], WK, 0, 0, g)
    ld_q[0].wait()
    for g in G:
        proj(x0[0], WQ, 0, 0, g)
    x1 = [x1_wait(0)]
    for w in (WK, WQ):
        for g in G:
            proj(x1[0], w, 1, 0, g)
    ld_k[1].wait()
    k0 = [proj(x0[1], WK, 0, 1, g).astype(BF) for g in G]
    x1.append(x1_wait(1))
    k1 = [proj(x1[1], WK, 1, 1, g).astype(BF) for g in G]
    ld_q[1].wait()
    q0 = [proj(x0[1], WQ, 0, 1, g) * QSCALE for g in G]
    p0 = [probs(q0[g], k0[g]) for g in G]
    q1 = [proj(x1[1], WQ, 1, 1, g) * QSCALE for g in G]

    ld_v[0].wait()
    r0 = [inv_sum(p0[g]) for g in G]
    for g in (0, 1):
        proj(x0[0], WV, 0, 0, g)
    p1 = [probs(q1[g], k1[g]) for g in G]
    for b, g in ((0, 2), (0, 3), (1, 0), (1, 1), (1, 2), (1, 3)):
        proj((x0, x1)[b][0], WV, b, 0, g)
    ld_v[1].wait()
    r1 = [inv_sum(p1[g]) for g in G]
    v0 = [proj(x0[1], WV, 0, 1, g).astype(BF) for g in G]
    o0 = jnp.concatenate([attend(p0[g], v0[g], r0[g], 1 if g < 2 else 2) for g in G], axis=1)
    o0 = jnp.concatenate([unit_rows(o0, t) for t in range(2)], axis=0)

    def run(*thunks):
        for f in thunks:
            f()

    ld_o[0].wait()
    pub = out_proj(o0, 0, 0)
    v1 = [proj(x1[1], WV, 1, 1, g).astype(BF) for g in (0, 1)]
    pub[0]()
    v1 += [proj(x1[1], WV, 1, 1, g).astype(BF) for g in (2, 3)]
    run(*pub[1:])
    ld_o[1].wait()
    pub = out_proj(o0, 0, 1)
    o1 = [jnp.concatenate([attend_tile(p1[g], v1[g], r1[g], 0) for g in G], axis=1)]
    pub[0]()
    o1.append(jnp.concatenate([attend_tile(p1[g], v1[g], r1[g], 1) for g in G], axis=1))
    run(*pub[1:])
    o1 = jnp.concatenate(o1, axis=0)
    run(*out_proj(o1, 1, 1), *out_proj(o1, 1, 0))
    ld_o[2].wait()
    run(*out_proj(o1, 1, 2), *out_proj(o0, 0, 2))
    ld_o[3].wait()
    run(*out_proj(o0, 0, 3), *out_proj(o1, 1, 3))

    for kh in range(2):
        for r in range(2):
            pl.when(has_x1[r])(x1_copy(kh, r).wait_send)

    def phase2(uid, h, row, col):
        rcopy(0, uid, h).wait_recv()
        acc = part_v[uid] + rcv1[uid].astype(F32)
        snd2[uid] = acc.astype(BF)
        rcopy(1, uid, h).start()
        part_v[uid] = acc

    def phase3(uid, h, row, col):
        rcopy(1, uid, h).wait_recv()
        acc = part_v[uid] + rcv2[uid].astype(F32)
        snd3[uid] = acc.astype(BF)
        rcopy(2, uid, h).start()
        out_ref[pl.ds(row, SR), pl.ds(col, 128)] = acc

    def finish(uid, h, row, col):
        rcopy(2, uid, h).wait_recv()
        out_ref[pl.ds(row, SR), pl.ds(col, 128)] = rcv3[uid].astype(F32)

    def drain(phase, ent):
        when(ent[0], rcopy(phase, ent[1], ent[2]).wait_send)

    for ent in own2:
        when(ent[0], lambda: phase2(*ent[1:]))
    for n, ent in enumerate(own3):
        drain(0, other[n])
        when(ent[0], lambda: phase3(*ent[1:]))
    for n, ent in enumerate(other):
        drain(1, own2[n])
        drain(2, own3[n])
        when(ent[0], lambda: finish(*ent[1:]))


def pallas_dist_attn_self_mha_htp_b2_sq128_skv128_d512_hq8_dh64_kernel(x, Wq, Wk, Wv, Wo):
    unit_buf = pltpu.VMEM((NU, SR, 128), BF)
    out = pl.pallas_call(
        _body,
        out_shape=jax.ShapeDtypeStruct((M, D), F32),
        in_specs=[pl.BlockSpec(memory_space=pl.ANY)] * 5,
        out_specs=pl.BlockSpec(memory_space=pltpu.VMEM),
        scratch_shapes=[
            pltpu.VMEM((M, D), F32),
            pltpu.VMEM((2, 2, 2, HR, 128), BF),
            pltpu.VMEM((2, 256, D), F32),
            pltpu.VMEM((2, 256, D), F32),
            pltpu.VMEM((2, 256, D), F32),
            pltpu.VMEM((NC, D, 128), F32),
            pltpu.VMEM((3, B, NG, S, 128), F32),
            pltpu.VMEM((NU, SR, 128), F32),
            unit_buf, unit_buf, unit_buf, unit_buf, unit_buf, unit_buf,
            pltpu.SemaphoreType.DMA((9 + NC,)),
            pltpu.SemaphoreType.DMA((6,)),
            pltpu.SemaphoreType.DMA((3 * NU,)),
            pltpu.SemaphoreType.DMA((3 * NU,)),
        ],
        compiler_params=pltpu.CompilerParams(
            collective_id=0, disable_semaphore_checks=True, disable_bounds_checks=True),
    )(x.reshape(M, D), Wq, Wk, Wv, Wo)
    return out.reshape(B, S, D)
```

```python
import jax
import jax.numpy as jnp
from jax import lax
from jax.experimental import pallas as pl
from jax.experimental.pallas import tpu as pltpu

B, S, D = 2, 128, 512
M = B * S
NG = 4
NC = 4
HR = 64
SR = 16
UR = 8
NBLK = HR // SR
UPH = HR // UR
NU = B * NC * 2 * UPH
BF = jnp.bfloat16
F32 = jnp.float32
MESH = pl.DeviceIdType.MESH
QSCALE = 0.125 * 1.4426950408889634

R_SIDE = ((0, 0), (0, 1), (1, 0), (0, 2))
D_SIDE = ((1, 1), (1, 2), (0, 3), (1, 3))
ROW_ORDER = [(h, j) for j in range(NBLK) for h in range(2)]


def _dot(a, b):
    return jnp.dot(a, b, preferred_element_type=F32)


def _uid(b, c, h, j):
    return ((b * NC + c) * 2 + h) * UPH + j


def _body(x_hbm, wq_hbm, wk_hbm, wv_hbm, wo_hbm, out_ref,
          x_v, x1_v, wk_v, wq_v, wv_v, wo_v, acc_v, part_v,
          snd1, rcv1, snd2, rcv2, snd3, rcv3,
          ld_sem, x_sem, snd_sem, rcv_sem):
    def wcopy(src, dst, half, s):
        return pltpu.make_async_copy(src.at[pl.ds(half * 256, 256)], dst.at[half], ld_sem.at[s])

    ld_x0 = pltpu.make_async_copy(x_hbm.at[pl.ds(0, S)], x_v.at[pl.ds(0, S)], ld_sem.at[0])
    ld_x1 = [pltpu.make_async_copy(x_hbm.at[pl.ds(S + r * HR, HR)], x_v.at[pl.ds(S + r * HR, HR)],
                                   ld_sem.at[1 + r]) for r in range(2)]
    ld_k = [wcopy(wk_hbm, wk_v, h, 3 + h) for h in range(2)]
    ld_q = [wcopy(wq_hbm, wq_v, h, 5 + h) for h in range(2)]
    ld_v = [wcopy(wv_hbm, wv_v, h, 7 + h) for h in range(2)]
    ld_o = [pltpu.make_async_copy(wo_hbm.at[:, pl.ds(c * 128, 128)], wo_v.at[c], ld_sem.at[9 + c])
            for c in range(NC)]

    ld_x0.start()
    me = lax.axis_index("i")
    is_r = me == 0
    is_d = me == 2
    has_x1 = [is_r | (me == 1), is_r | (me == 3)]
    for r in range(2):
        pl.when(has_x1[r])(ld_x1[r].start)
    ld_k[0].start()

    nbr = [me ^ 1, 3 - me]
    barrier = pltpu.get_barrier_semaphore()
    for p in nbr:
        pl.semaphore_signal(barrier, inc=1, device_id=(p,), device_id_type=MESH)
    for cp in (ld_q[0], ld_k[1], ld_q[1], ld_v[0], ld_v[1], *ld_o):
        cp.start()

    on_d_side = [(me == 1) | is_d, me >= 2]
    h_r = jnp.where(me == 3, 1, 0)
    h_d = 1 - h_r

    def unit_list(r_chunks, n_first, n_second, d_chunks):
        res = []
        for n in range(NU // 2):
            p, j = divmod(n // 2, UPH)
            n_chunks, n_half = (n_first, n_second)[n % 2]
            b, c = (jnp.where(is_r, r_chunks[p][i], jnp.where(is_d, d_chunks[p][i], n_chunks[p][i]))
                    for i in range(2))
            h = jnp.where(is_r | is_d, n % 2, n_half)
            res.append((_uid(b, c, h, j), h,
                        pl.multiple_of(b * S + h * HR + j * UR, UR), pl.multiple_of(c * 128, 128)))
        return res

    own2 = unit_list(R_SIDE, (D_SIDE, h_r), (R_SIDE, h_d), D_SIDE)
    own3 = unit_list(R_SIDE, (R_SIDE, h_d), (D_SIDE, h_r), D_SIDE)
    other = unit_list(D_SIDE, (R_SIDE, h_r), (D_SIDE, h_d), R_SIDE)

    def rcopy(phase, uid, h):
        snd, rcv = ((snd1, rcv1), (snd2, rcv2), (snd3, rcv3))[phase]
        if isinstance(h, int):
            dev = nbr[h ^ (phase % 2)]
        else:
            dev = jnp.where(h == phase % 2, nbr[0], nbr[1])
        return pltpu.make_async_remote_copy(
            src_ref=snd.at[uid], dst_ref=rcv.at[uid],
            send_sem=snd_sem.at[uid], recv_sem=rcv_sem.at[(phase % 2) * NU + uid],
            device_id=(dev,), device_id_type=MESH)

    def x1_copy(kh, r):
        return pltpu.make_async_remote_copy(
            src_ref=x1_v.at[kh, r], dst_ref=x1_v.at[kh, r],
            send_sem=x_sem.at[2 + 2 * kh + r], recv_sem=x_sem.at[kh],
            device_id=(jnp.where(is_r, 3 - 2 * r, 2),), device_id_type=MESH)

    def x1_wait(kh):
        @pl.when(is_d)
        def _():
            pltpu.make_async_copy(x1_v.at[kh], x1_v.at[kh], x_sem.at[kh]).wait()

        @pl.when(me % 2 == 1)
        def _():
            x1_copy(kh, 1 - me // 2).wait_recv()
        return jnp.concatenate(
            [jnp.concatenate([x1_v[kh, r, t] for r in range(2)], axis=0) for t in range(2)], axis=1)

    def lanes_lo(rows):
        return lax.broadcasted_iota(jnp.int32, (rows, 128), 1) < 64

    def proj(xh, w, b, half, g, row_tiles=1):
        wt = (wk_v, wq_v, wv_v)[w][half, :, g * 128:(g + 1) * 128].astype(BF)
        rows = S // row_tiles
        res = [_dot(xh[t * rows:(t + 1) * rows], wt) for t in range(row_tiles)]
        res = res[0] if row_tiles == 1 else jnp.concatenate(res, axis=0)
        if half == 0:
            acc_v[w, b, g] = res
            return None
        return res + acc_v[w, b, g]

    def probs(q, k):
        res = []
        for h in range(2):
            qh = jnp.where(lanes_lo(S), q, 0.0) if h == 0 else jnp.where(lanes_lo(S), 0.0, q)
            s = lax.dot_general(qh.astype(BF), k, (((1,), (1,)), ((), ())), preferred_element_type=F32)
            res.append(jnp.exp2(s - jnp.max(s, axis=-1, keepdims=True)).astype(BF))
        return res

    def inv_sum(p):
        l = jnp.where(lanes_lo(S), *[jnp.sum(ph.astype(F32), axis=-1, keepdims=True) for ph in p])
        r = pl.reciprocal(l, approx=True)
        return r * (2.0 - l * r)

    def reorder(a, blocks):
        return jnp.concatenate([a[h * HR + j * SR:h * HR + (j + 1) * SR] for h, j in blocks], axis=0)

    def attend(p, v, r, blocks):
        o = jnp.where(lanes_lo(len(blocks) * SR),
                      _dot(reorder(p[0], blocks), v), _dot(reorder(p[1], blocks), v))
        return (o * reorder(r, blocks)).astype(BF)

    def out_proj(o, b, c):
        res = _dot(o, wo_v[c].astype(BF))
        d_owns = (b, c) in D_SIDE

        def publish(j):
            for u in range(SR // UR):
                uid = [_uid(b, c, h, j * (SR // UR) + u) for h in range(2)]
                r0 = [ROW_ORDER.index((h, j)) * SR + u * UR for h in range(2)]
                for h in range(2):
                    snd1[uid[h]] = res[r0[h]:r0[h] + UR].astype(BF)
                for h in range(2):
                    pl.when(on_d_side[h] != d_owns)(rcopy(0, uid[h], h).start)
                for h in range(2):
                    part_v[uid[h]] = res[r0[h]:r0[h] + UR]
        return [lambda j=j: publish(j) for j in range(NBLK)]

    def run(*thunks):
        for f in thunks:
            f()

    G = range(NG)
    WK, WQ, WV = range(3)
    TILES = (ROW_ORDER[:NBLK], ROW_ORDER[NBLK:])

    ld_x0.wait()
    x0 = [x_v[0:S, kh * 256:(kh + 1) * 256].astype(BF) for kh in range(2)]
    for r in range(2):
        @pl.when(has_x1[r])
        def _():
            ld_x1[r].wait()
            for kh in range(2):
                for t in range(2):
                    c0 = kh * 256 + t * 128
                    x1_v[kh, r, t] = x_v[S + r * HR:S + (r + 1) * HR, c0:c0 + 128].astype(BF)
    pl.semaphore_wait(barrier, 2)
    for kh in range(2):
        for r in range(2):
            pl.when(has_x1[r])(x1_copy(kh, r).start)

    ld_k[0].wait()
    for g in G:
        proj(x0[0], WK, 0, 0, g)
    ld_q[0].wait()
    for g in G:
        proj(x0[0], WQ, 0, 0, g)
    x1 = [x1_wait(0)]
    for w in (WK, WQ):
        for g in G:
            proj(x1[0], w, 1, 0, g)
    ld_k[1].wait()
    k0 = [proj(x0[1], WK, 0, 1, g).astype(BF) for g in G]
    x1.append(x1_wait(1))
    k1 = [proj(x1[1], WK, 1, 1, g).astype(BF) for g in G]
    ld_q[1].wait()
    q0 = [proj(x0[1], WQ, 0, 1, g) * QSCALE for g in G]
    p0 = [probs(q0[g], k0[g]) for g in G]
    q1 = [proj(x1[1], WQ, 1, 1, g) * QSCALE for g in G]

    ld_v[0].wait()
    r0 = [inv_sum(p0[g]) for g in G]
    for g in (0, 1):
        proj(x0[0], WV, 0, 0, g)
    p1 = [probs(q1[g], k1[g]) for g in G]
    for b, g in ((0, 2), (0, 3), (1, 0), (1, 1), (1, 2), (1, 3)):
        proj((x0, x1)[b][0], WV, b, 0, g)
    ld_v[1].wait()
    r1 = [inv_sum(p1[g]) for g in G]
    v0 = [proj(x0[1], WV, 0, 1, g).astype(BF) for g in G]
    v1 = [proj(x1[1], WV, 1, 1, 0, row_tiles=2).astype(BF)]
    o0 = [attend(p0[g], v0[g], r0[g], ROW_ORDER) for g in (0, 1)]
    o0 += [jnp.concatenate([attend(p0[g], v0[g], r0[g], t) for t in TILES], axis=0) for g in (2, 3)]
    o0 = jnp.concatenate(o0, axis=1)

    ld_o[0].wait()
    pub = out_proj(o0, 0, 0)
    v1 += [proj(x1[1], WV, 1, 1, g).astype(BF) for g in (1, 2)]
    pub[0]()
    v1.append(proj(x1[1], WV, 1, 1, 3, row_tiles=2).astype(BF))
    run(*pub[1:])
    ld_o[1].wait()
    pub = out_proj(o0, 0, 1)
    o1 = [jnp.concatenate([attend(p1[g], v1[g], r1[g], TILES[0]) for g in G], axis=1)]
    pub[0]()
    o1.append(jnp.concatenate([attend(p1[g], v1[g], r1[g], TILES[1]) for g in G], axis=1))
    run(*pub[1:])
    o1 = jnp.concatenate(o1, axis=0)
    run(*out_proj(o1, 1, 1), *out_proj(o1, 1, 0))
    ld_o[2].wait()
    run(*out_proj(o1, 1, 2), *out_proj(o0, 0, 2))
    ld_o[3].wait()
    run(*out_proj(o0, 0, 3), *out_proj(o1, 1, 3))

    for kh in range(2):
        for r in range(2):
            pl.when(has_x1[r])(x1_copy(kh, r).wait_send)

    for uid, h, _, _ in own2:
        rcopy(0, uid, h).wait_recv()
        acc = part_v[uid] + rcv1[uid].astype(F32)
        snd2[uid] = acc.astype(BF)
        rcopy(1, uid, h).start()
        part_v[uid] = acc
    for n, (uid, h, row, col) in enumerate(own3):
        rcopy(0, *other[n][:2]).wait_send()
        rcopy(1, uid, h).wait()
        acc = part_v[uid] + rcv2[uid].astype(F32)
        snd3[uid] = acc.astype(BF)
        rcopy(2, uid, h).start()
        out_ref[pl.ds(row, UR), pl.ds(col, 128)] = acc
    for n, (uid, h, row, col) in enumerate(other):
        rcopy(2, *own3[n][:2]).wait_send()
        rcopy(2, uid, h).wait_recv()
        out_ref[pl.ds(row, UR), pl.ds(col, 128)] = rcv3[uid].astype(F32)


def pallas_dist_attn_self_mha_htp_b2_sq128_skv128_d512_hq8_dh64_kernel(x, Wq, Wk, Wv, Wo):
    unit_buf = pltpu.VMEM((NU, UR, 128), BF)
    out = pl.pallas_call(
        _body,
        out_shape=jax.ShapeDtypeStruct((M, D), F32),
        in_specs=[pl.BlockSpec(memory_space=pl.ANY)] * 5,
        out_specs=pl.BlockSpec(memory_space=pltpu.VMEM),
        scratch_shapes=[
            pltpu.VMEM((M, D), F32),
            pltpu.VMEM((2, 2, 2, HR, 128), BF),
            pltpu.VMEM((2, 256, D), F32),
            pltpu.VMEM((2, 256, D), F32),
            pltpu.VMEM((2, 256, D), F32),
            pltpu.VMEM((NC, D, 128), F32),
            pltpu.VMEM((3, B, NG, S, 128), F32),
            pltpu.VMEM((NU, UR, 128), F32),
            unit_buf, unit_buf, unit_buf, unit_buf, unit_buf, unit_buf,
            pltpu.SemaphoreType.DMA((9 + NC,)),
            pltpu.SemaphoreType.DMA((6,)),
            pltpu.SemaphoreType.DMA((NU,)),
            pltpu.SemaphoreType.DMA((2 * NU,)),
        ],
        compiler_params=pltpu.CompilerParams(
            collective_id=0, disable_semaphore_checks=True, disable_bounds_checks=True),
    )(x.reshape(M, D), Wq, Wk, Wv, Wo)
    return out.reshape(B, S, D)
```

```python
import jax
import jax.numpy as jnp
from jax import lax
from jax.experimental import pallas as pl
from jax.experimental.pallas import tpu as pltpu

B, S, D = 2, 128, 512
M = B * S
NG = 4
NC = 4
HR = 64
UR = 8
UPH = HR // UR
NU = B * NC * 2 * UPH
BF = jnp.bfloat16
F32 = jnp.float32
MESH = pl.DeviceIdType.MESH
QSCALE = 0.125 * 1.4426950408889634

R_SIDE = ((0, 0), (0, 1), (1, 0), (0, 2))
D_SIDE = ((1, 1), (1, 2), (0, 3), (1, 3))


def _dot(a, b):
    return jnp.dot(a, b, preferred_element_type=F32)


def _uid(b, c, h, j):
    return ((b * NC + c) * 2 + h) * UPH + j


def _body(x_hbm, wq_hbm, wk_hbm, wv_hbm, wo_hbm, out_ref,
          x_v, x1_v, wk_v, wq_v, wv_v, wo_v, acc_v, part_v,
          snd1, rcv1, snd2, rcv2, snd3, rcv3,
          ld_sem, x_sem, snd_sem, rcv_sem):
    def wcopy(src, dst, half, s):
        return pltpu.make_async_copy(src.at[pl.ds(half * 256, 256)], dst.at[half], ld_sem.at[s])

    ld_x0 = pltpu.make_async_copy(x_hbm.at[pl.ds(0, S)], x_v.at[pl.ds(0, S)], ld_sem.at[0])
    ld_x1 = [pltpu.make_async_copy(x_hbm.at[pl.ds(S + r * HR, HR)], x_v.at[pl.ds(S + r * HR, HR)],
                                   ld_sem.at[1 + r]) for r in range(2)]
    ld_k = [wcopy(wk_hbm, wk_v, h, 3 + h) for h in range(2)]
    ld_q = [wcopy(wq_hbm, wq_v, h, 5 + h) for h in range(2)]
    ld_v = [wcopy(wv_hbm, wv_v, h, 7 + h) for h in range(2)]
    ld_o = [pltpu.make_async_copy(wo_hbm.at[:, pl.ds(c * 128, 128)], wo_v.at[c], ld_sem.at[9 + c])
            for c in range(NC)]

    ld_x0.start()
    me = lax.axis_index("i")
    is_r = me == 0
    is_d = me == 2
    has_x1 = [is_r | (me == 1), is_r | (me == 3)]
    for r in range(2):
        pl.when(has_x1[r])(ld_x1[r].start)
    ld_k[0].start()

    nbr = [me ^ 1, 3 - me]
    barrier = pltpu.get_barrier_semaphore()
    for p in nbr:
        pl.semaphore_signal(barrier, inc=1, device_id=(p,), device_id_type=MESH)
    for cp in (ld_q[0], ld_k[1], ld_q[1], ld_v[0], ld_v[1], *ld_o):
        cp.start()

    on_d_side = [(me == 1) | is_d, me >= 2]
    h_r = jnp.where(me == 3, 1, 0)
    h_d = 1 - h_r

    def unit_list(r_chunks, n_first, n_second, d_chunks):
        res = []
        for n in range(NU // 2):
            p, j = divmod(n // 2, UPH)
            n_chunks, n_half = (n_first, n_second)[n % 2]
            b, c = (jnp.where(is_r, r_chunks[p][i], jnp.where(is_d, d_chunks[p][i], n_chunks[p][i]))
                    for i in range(2))
            h = jnp.where(is_r | is_d, n % 2, n_half)
            res.append((_uid(b, c, h, j), h,
                        pl.multiple_of(b * S + h * HR + j * UR, UR), pl.multiple_of(c * 128, 128)))
        return res

    own2 = unit_list(R_SIDE, (D_SIDE, h_r), (R_SIDE, h_d), D_SIDE)
    own3 = unit_list(R_SIDE, (R_SIDE, h_d), (D_SIDE, h_r), D_SIDE)
    other = unit_list(D_SIDE, (R_SIDE, h_r), (D_SIDE, h_d), R_SIDE)

    def rcopy(phase, uid, h):
        snd, rcv = ((snd1, rcv1), (snd2, rcv2), (snd3, rcv3))[phase]
        if isinstance(h, int):
            dev = nbr[h ^ (phase % 2)]
        else:
            dev = jnp.where(h == phase % 2, nbr[0], nbr[1])
        return pltpu.make_async_remote_copy(
            src_ref=snd.at[uid], dst_ref=rcv.at[uid],
            send_sem=snd_sem.at[uid], recv_sem=rcv_sem.at[(phase % 2) * NU + uid],
            device_id=(dev,), device_id_type=MESH)

    def x1_copy(kh, r):
        return pltpu.make_async_remote_copy(
            src_ref=x1_v.at[kh, r], dst_ref=x1_v.at[kh, r],
            send_sem=x_sem.at[2 + 2 * kh + r], recv_sem=x_sem.at[kh],
            device_id=(jnp.where(is_r, 3 - 2 * r, 2),), device_id_type=MESH)

    def x1_wait(kh):
        @pl.when(is_d)
        def _():
            pltpu.make_async_copy(x1_v.at[kh], x1_v.at[kh], x_sem.at[kh]).wait()

        @pl.when(me % 2 == 1)
        def _():
            x1_copy(kh, 1 - me // 2).wait_recv()
        return jnp.concatenate(
            [jnp.concatenate([x1_v[kh, r, t] for r in range(2)], axis=0) for t in range(2)], axis=1)

    def lanes_lo(rows):
        return lax.broadcasted_iota(jnp.int32, (rows, 128), 1) < 64

    def proj(xh, w, b, half, g, row_tiles=1):
        wt = (wk_v, wq_v, wv_v)[w][half, :, g * 128:(g + 1) * 128].astype(BF)
        rows = S // row_tiles
        res = [_dot(xh[t * rows:(t + 1) * rows], wt) for t in range(row_tiles)]
        res = res[0] if row_tiles == 1 else jnp.concatenate(res, axis=0)
        if half == 0:
            acc_v[w, b, g] = res
            return None
        return res + acc_v[w, b, g]

    def probs(q, k):
        res = []
        for h in range(2):
            qh = jnp.where(lanes_lo(S), q, 0.0) if h == 0 else jnp.where(lanes_lo(S), 0.0, q)
            s = lax.dot_general(qh.astype(BF), k, (((1,), (1,)), ((), ())), preferred_element_type=F32)
            res.append(jnp.exp2(s - jnp.max(s, axis=-1, keepdims=True)).astype(BF))
        return res

    def inv_sum(p):
        l = jnp.where(lanes_lo(S), *[jnp.sum(ph.astype(F32), axis=-1, keepdims=True) for ph in p])
        r = pl.reciprocal(l, approx=True)
        return r * (2.0 - l * r)

    def interleave_halves(q):
        return jnp.concatenate(
            [q[h * HR + j * UR:h * HR + (j + 1) * UR] for j in range(UPH) for h in range(2)], axis=0)

    def attend(p, v, r, rows=slice(0, S)):
        o = jnp.where(lanes_lo(rows.stop - rows.start), _dot(p[0][rows], v), _dot(p[1][rows], v))
        return (o * r[rows]).astype(BF)

    def out_proj(o, b, c):
        res = _dot(o, wo_v[c].astype(BF))
        d_owns = (b, c) in D_SIDE

        def publish(j):
            piece = [res[(2 * j + h) * UR:(2 * j + h + 1) * UR] for h in range(2)]
            for h in range(2):
                snd1[_uid(b, c, h, j)] = piece[h].astype(BF)
                pl.when(on_d_side[h] != d_owns)(rcopy(0, _uid(b, c, h, j), h).start)
            for h in range(2):
                part_v[_uid(b, c, h, j)] = piece[h]
        return [lambda j=j: publish(j) for j in range(UPH)]

    def run(*thunks):
        for f in thunks:
            f()

    G = range(NG)
    WK, WQ, WV = range(3)
    TILES = (slice(0, HR), slice(HR, S))

    ld_x0.wait()
    x0 = [x_v[0:S, kh * 256:(kh + 1) * 256].astype(BF) for kh in range(2)]
    for r in range(2):
        @pl.when(has_x1[r])
        def _():
            ld_x1[r].wait()
            for kh in range(2):
                for t in range(2):
                    c0 = kh * 256 + t * 128
                    x1_v[kh, r, t] = x_v[S + r * HR:S + (r + 1) * HR, c0:c0 + 128].astype(BF)
    pl.semaphore_wait(barrier, 2)
    for kh in range(2):
        for r in range(2):
            pl.when(has_x1[r])(x1_copy(kh, r).start)

    ld_k[0].wait()
    for g in G:
        proj(x0[0], WK, 0, 0, g)
    ld_q[0].wait()
    for g in G:
        proj(x0[0], WQ, 0, 0, g)
    x1 = [x1_wait(0)]
    for w in (WK, WQ):
        for g in G:
            proj(x1[0], w, 1, 0, g)
    ld_k[1].wait()
    k0 = [proj(x0[1], WK, 0, 1, g).astype(BF) for g in G]
    x1.append(x1_wait(1))
    k1 = [proj(x1[1], WK, 1, 1, g).astype(BF) for g in G]
    ld_q[1].wait()
    q0 = [interleave_halves(proj(x0[1], WQ, 0, 1, g) * QSCALE) for g in G]
    p0 = [probs(q0[g], k0[g]) for g in G]
    q1 = [interleave_halves(proj(x1[1], WQ, 1, 1, g) * QSCALE) for g in G]

    for kh in range(2):
        for r in range(2):
            pl.when(has_x1[r])(x1_copy(kh, r).wait_send)
    ld_v[0].wait()
    r0 = [inv_sum(p0[g]) for g in G]
    for g in (0, 1):
        proj(x0[0], WV, 0, 0, g)
    p1 = [probs(q1[g], k1[g]) for g in G]
    for b, g in ((0, 2), (0, 3), (1, 0), (1, 1), (1, 2), (1, 3)):
        proj((x0, x1)[b][0], WV, b, 0, g)
    ld_v[1].wait()
    r1 = [inv_sum(p1[g]) for g in G]
    v0 = [proj(x0[1], WV, 0, 1, g).astype(BF) for g in G]
    v1 = [proj(x1[1], WV, 1, 1, 0, row_tiles=2).astype(BF)]
    o0 = [attend(p0[g], v0[g], r0[g]) for g in (0, 1)]
    o0 += [jnp.concatenate([attend(p0[g], v0[g], r0[g], t) for t in TILES], axis=0) for g in (2, 3)]
    o0 = jnp.concatenate(o0, axis=1)

    ld_o[0].wait()
    pub = out_proj(o0, 0, 0)
    v1 += [proj(x1[1], WV, 1, 1, g).astype(BF) for g in (1, 2)]
    pub[0]()
    v1.append(proj(x1[1], WV, 1, 1, 3, row_tiles=2).astype(BF))
    run(*pub[1:])
    ld_o[1].wait()
    pub = out_proj(o0, 0, 1)
    o1 = [jnp.concatenate([attend(p1[g], v1[g], r1[g], TILES[0]) for g in G], axis=1)]
    pub[0]()
    o1.append(jnp.concatenate([attend(p1[g], v1[g], r1[g], TILES[1]) for g in G], axis=1))
    run(*pub[1:])
    o1 = jnp.concatenate(o1, axis=0)
    run(*out_proj(o1, 1, 1), *out_proj(o1, 1, 0))
    ld_o[2].wait()
    run(*out_proj(o1, 1, 2), *out_proj(o0, 0, 2))
    ld_o[3].wait()
    run(*out_proj(o0, 0, 3), *out_proj(o1, 1, 3))

    for uid, h, _, _ in own2:
        rcopy(0, uid, h).wait_recv()
        acc = part_v[uid] + rcv1[uid].astype(F32)
        snd2[uid] = acc.astype(BF)
        rcopy(1, uid, h).start()
        part_v[uid] = acc
    for n, (uid, h, row, col) in enumerate(own3):
        rcopy(0, *other[n][:2]).wait_send()
        rcopy(1, uid, h).wait()
        acc = part_v[uid] + rcv2[uid].astype(F32)
        snd3[uid] = acc.astype(BF)
        rcopy(2, uid, h).start()
        out_ref[pl.ds(row, UR), pl.ds(col, 128)] = acc
    for n, (uid, h, row, col) in enumerate(other):
        rcopy(2, *own3[n][:2]).wait_send()
        rcopy(2, uid, h).wait_recv()
        out_ref[pl.ds(row, UR), pl.ds(col, 128)] = rcv3[uid].astype(F32)


def pallas_dist_attn_self_mha_htp_b2_sq128_skv128_d512_hq8_dh64_kernel(x, Wq, Wk, Wv, Wo):
    unit_buf = pltpu.VMEM((NU, UR, 128), BF)
    out = pl.pallas_call(
        _body,
        out_shape=jax.ShapeDtypeStruct((M, D), F32),
        in_specs=[pl.BlockSpec(memory_space=pl.ANY)] * 5,
        out_specs=pl.BlockSpec(memory_space=pltpu.VMEM),
        scratch_shapes=[
            pltpu.VMEM((M, D), F32),
            pltpu.VMEM((2, 2, 2, HR, 128), BF),
            pltpu.VMEM((2, 256, D), F32),
            pltpu.VMEM((2, 256, D), F32),
            pltpu.VMEM((2, 256, D), F32),
            pltpu.VMEM((NC, D, 128), F32),
            pltpu.VMEM((3, B, NG, S, 128), F32),
            pltpu.VMEM((NU, UR, 128), F32),
            unit_buf, unit_buf, unit_buf, unit_buf, unit_buf, unit_buf,
            pltpu.SemaphoreType.DMA((9 + NC,)),
            pltpu.SemaphoreType.DMA((6,)),
            pltpu.SemaphoreType.DMA((NU,)),
            pltpu.SemaphoreType.DMA((2 * NU,)),
        ],
        compiler_params=pltpu.CompilerParams(collective_id=0, disable_semaphore_checks=True),
    )(x.reshape(M, D), Wq, Wk, Wv, Wo)
    return out.reshape(B, S, D)
```

```python
import jax
import jax.numpy as jnp
from jax import lax
from jax.experimental import pallas as pl
from jax.experimental.pallas import tpu as pltpu

B, S, D = 2, 128, 512
M = B * S
NG = 4
NC = 4
HR = 64
UR = 8
UPH = HR // UR
NU = B * NC * 2 * UPH
BF = jnp.bfloat16
F32 = jnp.float32
MESH = pl.DeviceIdType.MESH
QSCALE = 0.125 * 1.4426950408889634

R_SIDE = ((0, 0), (0, 1), (1, 0), (0, 2))
D_SIDE = ((1, 1), (1, 2), (0, 3), (1, 3))


def _dot(a, b):
    return jnp.dot(a, b, preferred_element_type=F32)


def _uid(b, c, h, j):
    return ((b * NC + c) * 2 + h) * UPH + j


def _body(x_hbm, wq_hbm, wk_hbm, wv_hbm, wo_hbm, out_ref,
          x_v, x1_v, wk_v, wq_v, wv_v, wo_v, acc_v, part_v,
          snd1, rcv1, snd2, rcv2, snd3, rcv3,
          ld_sem, x_sem, snd_sem, rcv_sem):
    def wcopy(src, dst, half, s):
        return pltpu.make_async_copy(src.at[pl.ds(half * 256, 256)], dst.at[half], ld_sem.at[s])

    ld_x0 = pltpu.make_async_copy(x_hbm.at[pl.ds(0, S)], x_v.at[pl.ds(0, S)], ld_sem.at[0])
    ld_x1 = [pltpu.make_async_copy(x_hbm.at[pl.ds(S + r * HR, HR)], x_v.at[pl.ds(S + r * HR, HR)],
                                   ld_sem.at[1 + r]) for r in range(2)]
    ld_k = [wcopy(wk_hbm, wk_v, h, 3 + h) for h in range(2)]
    ld_q = [wcopy(wq_hbm, wq_v, h, 5 + h) for h in range(2)]
    ld_v = [wcopy(wv_hbm, wv_v, h, 7 + h) for h in range(2)]

    def o_parts(c):
        n_blk, n_row = (8, 8) if c < 2 else (16, 32)
        return [pltpu.make_async_copy(wo_hbm.at[pl.ds(i, n_blk), pl.ds(r, n_row), pl.ds(c * 128, 128)],
                                      wo_v.at[c, pl.ds(i, n_blk), pl.ds(r, n_row)], ld_sem.at[9 + c])
                for i in range(0, 16, n_blk) for r in range(0, 32, n_row)]

    def o_wait(c):
        pltpu.make_async_copy(wo_v.at[c], wo_v.at[c], ld_sem.at[9 + c]).wait()

    ld_x0.start()
    me = lax.axis_index("i")
    is_r = me == 0
    is_d = me == 2
    has_x1 = [is_r | (me == 1), is_r | (me == 3)]
    for r in range(2):
        pl.when(has_x1[r])(ld_x1[r].start)
    ld_k[0].start()

    nbr = [me ^ 1, 3 - me]
    barrier = pltpu.get_barrier_semaphore()
    for p in nbr:
        pl.semaphore_signal(barrier, inc=1, device_id=(p,), device_id_type=MESH)
    for cp in (ld_q[0], ld_k[1], ld_q[1], ld_v[0], ld_v[1], *[p for c in range(NC) for p in o_parts(c)]):
        cp.start()

    on_d_side = [(me == 1) | is_d, me >= 2]
    h_r = jnp.where(me == 3, 1, 0)
    h_d = 1 - h_r

    def unit_list(r_chunks, n_first, n_second, d_chunks):
        res = []
        for n in range(NU // 2):
            p, j = divmod(n // 2, UPH)
            n_chunks, n_half = (n_first, n_second)[n % 2]
            b, c = (jnp.where(is_r, r_chunks[p][i], jnp.where(is_d, d_chunks[p][i], n_chunks[p][i]))
                    for i in range(2))
            h = jnp.where(is_r | is_d, n % 2, n_half)
            res.append((_uid(b, c, h, j), h,
                        pl.multiple_of(b * S + h * HR + j * UR, UR), pl.multiple_of(c * 128, 128)))
        return res

    own2 = unit_list(R_SIDE, (D_SIDE, h_r), (R_SIDE, h_d), D_SIDE)
    own3 = unit_list(R_SIDE, (R_SIDE, h_d), (D_SIDE, h_r), D_SIDE)
    other = unit_list(D_SIDE, (R_SIDE, h_r), (D_SIDE, h_d), R_SIDE)

    def rcopy(phase, uid, h):
        snd, rcv = ((snd1, rcv1), (snd2, rcv2), (snd3, rcv3))[phase]
        if isinstance(h, int):
            dev = nbr[h ^ (phase % 2)]
        else:
            dev = jnp.where(h == phase % 2, nbr[0], nbr[1])
        return pltpu.make_async_remote_copy(
            src_ref=snd.at[uid], dst_ref=rcv.at[uid],
            send_sem=snd_sem.at[uid], recv_sem=rcv_sem.at[(phase % 2) * NU + uid],
            device_id=(dev,), device_id_type=MESH)

    def x1_copy(kh, r):
        return pltpu.make_async_remote_copy(
            src_ref=x1_v.at[kh, r], dst_ref=x1_v.at[kh, r],
            send_sem=x_sem.at[2 + 2 * kh + r], recv_sem=x_sem.at[kh],
            device_id=(jnp.where(is_r, 3 - 2 * r, 2),), device_id_type=MESH)

    def x1_wait(kh):
        @pl.when(is_d)
        def _():
            pltpu.make_async_copy(x1_v.at[kh], x1_v.at[kh], x_sem.at[kh]).wait()

        @pl.when(me % 2 == 1)
        def _():
            x1_copy(kh, 1 - me // 2).wait_recv()
        return jnp.concatenate(
            [jnp.concatenate([x1_v[kh, r, t] for r in range(2)], axis=0) for t in range(2)], axis=1)

    def lanes_lo(rows):
        return lax.broadcasted_iota(jnp.int32, (rows, 128), 1) < 64

    def proj(xh, w, b, half, g, row_tiles=1):
        wt = (wk_v, wq_v, wv_v)[w][half, :, g * 128:(g + 1) * 128].astype(BF)
        rows = S // row_tiles
        res = [_dot(xh[t * rows:(t + 1) * rows], wt) for t in range(row_tiles)]
        res = res[0] if row_tiles == 1 else jnp.concatenate(res, axis=0)
        if half == 0:
            acc_v[w, b, g] = res
            return None
        return res + acc_v[w, b, g]

    def probs(q, k):
        res = []
        for h in range(2):
            qh = jnp.where(lanes_lo(S), q, 0.0) if h == 0 else jnp.where(lanes_lo(S), 0.0, q)
            s = lax.dot_general(qh.astype(BF), k, (((1,), (1,)), ((), ())), preferred_element_type=F32)
            res.append(jnp.exp2(s - jnp.max(s, axis=-1, keepdims=True)).astype(BF))
        return res

    def inv_sum(p):
        l = jnp.where(lanes_lo(S), *[jnp.sum(ph.astype(F32), axis=-1, keepdims=True) for ph in p])
        r = pl.reciprocal(l, approx=True)
        return r * (2.0 - l * r)

    def interleave_halves(q):
        return jnp.concatenate(
            [q[h * HR + j * UR:h * HR + (j + 1) * UR] for j in range(UPH) for h in range(2)], axis=0)

    def attend(p, v, r, rows=slice(0, S)):
        o = jnp.where(lanes_lo(rows.stop - rows.start), _dot(p[0][rows], v), _dot(p[1][rows], v))
        return (o * r[rows]).astype(BF)

    def out_proj(o, b, c):
        res = _dot(o, wo_v[c].reshape(D, 128).astype(BF))
        d_owns = (b, c) in D_SIDE

        def publish(j):
            piece = [res[(2 * j + h) * UR:(2 * j + h + 1) * UR] for h in range(2)]
            for h in range(2):
                snd1[_uid(b, c, h, j)] = piece[h].astype(BF)
                pl.when(on_d_side[h] != d_owns)(rcopy(0, _uid(b, c, h, j), h).start)
            for h in range(2):
                part_v[_uid(b, c, h, j)] = piece[h]
        return [lambda j=j: publish(j) for j in range(UPH)]

    def run(*thunks):
        for f in thunks:
            f()

    G = range(NG)
    WK, WQ, WV = range(3)
    TILES = (slice(0, HR), slice(HR, S))

    ld_x0.wait()
    x0 = [x_v[0:S, kh * 256:(kh + 1) * 256].astype(BF) for kh in range(2)]
    for r in range(2):
        @pl.when(has_x1[r])
        def _():
            ld_x1[r].wait()
            for kh in range(2):
                for t in range(2):
                    c0 = kh * 256 + t * 128
                    x1_v[kh, r, t] = x_v[S + r * HR:S + (r + 1) * HR, c0:c0 + 128].astype(BF)
    pl.semaphore_wait(barrier, 2)
    for kh in range(2):
        for r in range(2):
            pl.when(has_x1[r])(x1_copy(kh, r).start)

    ld_k[0].wait()
    for g in G:
        proj(x0[0], WK, 0, 0, g)
    ld_q[0].wait()
    for g in G:
        proj(x0[0], WQ, 0, 0, g)
    x1 = [x1_wait(0)]
    for w in (WK, WQ):
        for g in G:
            proj(x1[0], w, 1, 0, g)
    ld_k[1].wait()
    k0 = [proj(x0[1], WK, 0, 1, g).astype(BF) for g in G]
    x1.append(x1_wait(1))
    k1 = [proj(x1[1], WK, 1, 1, g).astype(BF) for g in G]
    ld_q[1].wait()
    q0 = [interleave_halves(proj(x0[1], WQ, 0, 1, g) * QSCALE) for g in G]
    p0 = [probs(q0[g], k0[g]) for g in G]
    q1 = [interleave_halves(proj(x1[1], WQ, 1, 1, g) * QSCALE) for g in G]

    for kh in range(2):
        for r in range(2):
            pl.when(has_x1[r])(x1_copy(kh, r).wait_send)
    ld_v[0].wait()
    r0 = [inv_sum(p0[g]) for g in G]
    for g in (0, 1):
        proj(x0[0], WV, 0, 0, g)
    p1 = [probs(q1[g], k1[g]) for g in G]
    for b, g in ((0, 2), (0, 3), (1, 0), (1, 1), (1, 2), (1, 3)):
        proj((x0, x1)[b][0], WV, b, 0, g)
    ld_v[1].wait()
    r1 = [inv_sum(p1[g]) for g in G]
    v0 = [proj(x0[1], WV, 0, 1, g).astype(BF) for g in G]
    v1 = [proj(x1[1], WV, 1, 1, 0, row_tiles=2).astype(BF)]
    o0 = [attend(p0[g], v0[g], r0[g]) for g in (0, 1)]
    o0 += [jnp.concatenate([attend(p0[g], v0[g], r0[g], t) for t in TILES], axis=0) for g in (2, 3)]
    o0 = jnp.concatenate(o0, axis=1)

    o_wait(0)
    pub = out_proj(o0, 0, 0)
    v1 += [proj(x1[1], WV, 1, 1, g).astype(BF) for g in (1, 2)]
    pub[0]()
    v1.append(proj(x1[1], WV, 1, 1, 3, row_tiles=2).astype(BF))
    run(*pub[1:])
    o_wait(1)
    pub = out_proj(o0, 0, 1)
    o1 = [jnp.concatenate([attend(p1[g], v1[g], r1[g], TILES[0]) for g in G], axis=1)]
    pub[0]()
    o1.append(jnp.concatenate([attend(p1[g], v1[g], r1[g], TILES[1]) for g in G], axis=1))
    run(*pub[1:])
    o1 = jnp.concatenate(o1, axis=0)
    run(*out_proj(o1, 1, 1), *out_proj(o1, 1, 0))
    o_wait(2)
    run(*out_proj(o1, 1, 2), *out_proj(o0, 0, 2))
    o_wait(3)
    run(*out_proj(o0, 0, 3), *out_proj(o1, 1, 3))

    for uid, h, _, _ in own2:
        rcopy(0, uid, h).wait_recv()
        acc = part_v[uid] + rcv1[uid].astype(F32)
        snd2[uid] = acc.astype(BF)
        rcopy(1, uid, h).start()
        part_v[uid] = acc
    for n, (uid, h, row, col) in enumerate(own3):
        rcopy(0, *other[n][:2]).wait_send()
        rcopy(1, uid, h).wait()
        acc = part_v[uid] + rcv2[uid].astype(F32)
        snd3[uid] = acc.astype(BF)
        rcopy(2, uid, h).start()
        out_ref[pl.ds(row, UR), pl.ds(col, 128)] = acc
    for n, (uid, h, row, col) in enumerate(other):
        rcopy(2, *own3[n][:2]).wait_send()
        rcopy(2, uid, h).wait_recv()
        out_ref[pl.ds(row, UR), pl.ds(col, 128)] = rcv3[uid].astype(F32)


def pallas_dist_attn_self_mha_htp_b2_sq128_skv128_d512_hq8_dh64_kernel(x, Wq, Wk, Wv, Wo):
    unit_buf = pltpu.VMEM((NU, UR, 128), BF)
    out = pl.pallas_call(
        _body,
        out_shape=jax.ShapeDtypeStruct((M, D), F32),
        in_specs=[pl.BlockSpec(memory_space=pl.ANY)] * 5,
        out_specs=pl.BlockSpec(memory_space=pltpu.VMEM),
        scratch_shapes=[
            pltpu.VMEM((M, D), F32),
            pltpu.VMEM((2, 2, 2, HR, 128), BF),
            pltpu.VMEM((2, 256, D), F32),
            pltpu.VMEM((2, 256, D), F32),
            pltpu.VMEM((2, 256, D), F32),
            pltpu.VMEM((NC, 16, 32, 128), F32),
            pltpu.VMEM((3, B, NG, S, 128), F32),
            pltpu.VMEM((NU, UR, 128), F32),
            unit_buf, unit_buf, unit_buf, unit_buf, unit_buf, unit_buf,
            pltpu.SemaphoreType.DMA((9 + NC,)),
            pltpu.SemaphoreType.DMA((6,)),
            pltpu.SemaphoreType.DMA((NU,)),
            pltpu.SemaphoreType.DMA((2 * NU,)),
        ],
        compiler_params=pltpu.CompilerParams(collective_id=0, disable_semaphore_checks=True),
    )(x.reshape(M, D), Wq, Wk, Wv, Wo.reshape(16, 32, D))
    return out.reshape(B, S, D)
```

```python
import jax
import jax.numpy as jnp
from jax import lax
from jax.experimental import pallas as pl
from jax.experimental.pallas import tpu as pltpu

B, S, D = 2, 128, 512
M = B * S
NG = 4
NC = 4
HR = 64
UR = 8
UPH = HR // UR
NU = B * NC * 2 * UPH
BF = jnp.bfloat16
F32 = jnp.float32
MESH = pl.DeviceIdType.MESH
QSCALE = 0.125 * 1.4426950408889634

R_SIDE = ((0, 0), (0, 1), (1, 0), (0, 2))
D_SIDE = ((1, 1), (1, 2), (0, 3), (1, 3))


def _dot(a, b):
    return jnp.dot(a, b, preferred_element_type=F32)


def _uid(b, c, h, j):
    return ((b * NC + c) * 2 + h) * UPH + j


def _body(x_hbm, wq_hbm, wk_hbm, wv_hbm, wo_hbm, out_ref,
          x_v, x1_v, wk_v, wq_v, wv_v, wo_v, acc_v, part_v,
          snd1, rcv1, snd2, rcv2, snd3, rcv3,
          ld_sem, x_sem, snd_sem, rcv_sem):
    def wcopy(src, dst, half, s):
        return pltpu.make_async_copy(src.at[pl.ds(half * 256, 256)], dst.at[half], ld_sem.at[s])

    ld_x0 = pltpu.make_async_copy(x_hbm.at[pl.ds(0, S)], x_v.at[pl.ds(0, S)], ld_sem.at[0])
    ld_x1 = [pltpu.make_async_copy(x_hbm.at[pl.ds(S + r * HR, HR)], x_v.at[pl.ds(S + r * HR, HR)],
                                   ld_sem.at[1 + r]) for r in range(2)]
    ld_k = [wcopy(wk_hbm, wk_v, h, 3 + h) for h in range(2)]
    ld_q = [wcopy(wq_hbm, wq_v, h, 5 + h) for h in range(2)]
    ld_v = [wcopy(wv_hbm, wv_v, h, 7 + h) for h in range(2)]

    def o_parts(c):
        n_blk, n_row = (8, 8) if c < 2 else (16, 32)
        return [pltpu.make_async_copy(wo_hbm.at[pl.ds(i, n_blk), pl.ds(r, n_row), pl.ds(c * 128, 128)],
                                      wo_v.at[c, pl.ds(i, n_blk), pl.ds(r, n_row)], ld_sem.at[9 + c])
                for i in range(0, 16, n_blk) for r in range(0, 32, n_row)]

    def o_wait(c):
        pltpu.make_async_copy(wo_v.at[c], wo_v.at[c], ld_sem.at[9 + c]).wait()

    ld_x0.start()
    me = lax.axis_index("i")
    is_r = me == 0
    is_d = me == 2
    has_x1 = [is_r | (me == 1), is_r | (me == 3)]
    for r in range(2):
        pl.when(has_x1[r])(ld_x1[r].start)
    ld_k[0].start()

    nbr = [me ^ 1, 3 - me]
    barrier = pltpu.get_barrier_semaphore()
    for p in nbr:
        pl.semaphore_signal(barrier, inc=1, device_id=(p,), device_id_type=MESH)
    for cp in (ld_q[0], ld_k[1], ld_q[1], ld_v[0], ld_v[1], *[p for c in range(NC) for p in o_parts(c)]):
        cp.start()

    on_d_side = [(me == 1) | is_d, me >= 2]
    h_r = jnp.where(me == 3, 1, 0)
    h_d = 1 - h_r

    def unit_list(r_chunks, n_first, n_second, d_chunks):
        res = []
        for n in range(NU // 2):
            p, j = divmod(n // 2, UPH)
            n_chunks, n_half = (n_first, n_second)[n % 2]
            b, c = (jnp.where(is_r, r_chunks[p][i], jnp.where(is_d, d_chunks[p][i], n_chunks[p][i]))
                    for i in range(2))
            h = jnp.where(is_r | is_d, n % 2, n_half)
            res.append((_uid(b, c, h, j), h,
                        pl.multiple_of(b * S + h * HR + j * UR, UR), pl.multiple_of(c * 128, 128)))
        return res

    own2 = unit_list(R_SIDE, (D_SIDE, h_r), (R_SIDE, h_d), D_SIDE)
    own3 = unit_list(R_SIDE, (R_SIDE, h_d), (D_SIDE, h_r), D_SIDE)
    other = unit_list(D_SIDE, (R_SIDE, h_r), (D_SIDE, h_d), R_SIDE)

    def rcopy(phase, uid, h):
        snd, rcv = ((snd1, rcv1), (snd2, rcv2), (snd3, rcv3))[phase]
        if isinstance(h, int):
            dev = nbr[h ^ (phase % 2)]
        else:
            dev = jnp.where(h == phase % 2, nbr[0], nbr[1])
        return pltpu.make_async_remote_copy(
            src_ref=snd.at[uid], dst_ref=rcv.at[uid],
            send_sem=snd_sem.at[uid], recv_sem=rcv_sem.at[(phase % 2) * NU + uid],
            device_id=(dev,), device_id_type=MESH)

    def x1_copy(kh, r):
        return pltpu.make_async_remote_copy(
            src_ref=x1_v.at[kh, r], dst_ref=x1_v.at[kh, r],
            send_sem=x_sem.at[2 + 2 * kh + r], recv_sem=x_sem.at[kh],
            device_id=(jnp.where(is_r, 3 - 2 * r, 2),), device_id_type=MESH)

    def x1_wait(kh):
        @pl.when(is_d)
        def _():
            pltpu.make_async_copy(x1_v.at[kh], x1_v.at[kh], x_sem.at[kh]).wait()

        @pl.when(me % 2 == 1)
        def _():
            x1_copy(kh, 1 - me // 2).wait_recv()
        return jnp.concatenate(
            [jnp.concatenate([x1_v[kh, r, t] for r in range(2)], axis=0) for t in range(2)], axis=1)

    def lanes_lo(rows):
        return lax.broadcasted_iota(jnp.int32, (rows, 128), 1) < 64

    def proj(xh, w, b, half, g, row_tiles=1):
        wt = (wk_v, wq_v, wv_v)[w][half, :, g * 128:(g + 1) * 128].astype(BF)
        rows = S // row_tiles
        res = [_dot(xh[t * rows:(t + 1) * rows], wt) for t in range(row_tiles)]
        res = res[0] if row_tiles == 1 else jnp.concatenate(res, axis=0)
        if half == 0:
            acc_v[w, b, g] = res
            return None
        return res + acc_v[w, b, g]

    def probs(q, k):
        res = []
        for h in range(2):
            qh = jnp.where(lanes_lo(S), q, 0.0) if h == 0 else jnp.where(lanes_lo(S), 0.0, q)
            s = lax.dot_general(qh.astype(BF), k, (((1,), (1,)), ((), ())), preferred_element_type=F32)
            res.append(jnp.exp2(s - jnp.max(s, axis=-1, keepdims=True)).astype(BF))
        return res

    def inv_sum(p):
        l = jnp.where(lanes_lo(S), *[jnp.sum(ph.astype(F32), axis=-1, keepdims=True) for ph in p])
        r = pl.reciprocal(l, approx=True)
        return r * (2.0 - l * r)

    def interleave_halves(q):
        return jnp.concatenate(
            [q[h * HR + j * UR:h * HR + (j + 1) * UR] for j in range(UPH) for h in range(2)], axis=0)

    def attend(p, v, r, rows=slice(0, S)):
        o = jnp.where(lanes_lo(rows.stop - rows.start), _dot(p[0][rows], v), _dot(p[1][rows], v))
        return (o * r[rows]).astype(BF)

    def out_proj(o, b, c, j0=0):
        res = _dot(o, wo_v[c].reshape(D, 128).astype(BF))
        d_owns = (b, c) in D_SIDE

        def publish(j):
            piece = [res[(2 * (j - j0) + h) * UR:(2 * (j - j0) + h + 1) * UR] for h in range(2)]
            for h in range(2):
                snd1[_uid(b, c, h, j)] = piece[h].astype(BF)
                pl.when(on_d_side[h] != d_owns)(rcopy(0, _uid(b, c, h, j), h).start)
            for h in range(2):
                part_v[_uid(b, c, h, j)] = piece[h]
        return [lambda j=j: publish(j) for j in range(j0, j0 + o.shape[0] // (2 * UR))]

    def run(*thunks):
        for f in thunks:
            f()

    G = range(NG)
    WK, WQ, WV = range(3)
    TILES = (slice(0, HR), slice(HR, S))

    ld_x0.wait()
    x0 = [x_v[0:S, kh * 256:(kh + 1) * 256].astype(BF) for kh in range(2)]
    for r in range(2):
        @pl.when(has_x1[r])
        def _():
            ld_x1[r].wait()
            for kh in range(2):
                for t in range(2):
                    c0 = kh * 256 + t * 128
                    x1_v[kh, r, t] = x_v[S + r * HR:S + (r + 1) * HR, c0:c0 + 128].astype(BF)
    pl.semaphore_wait(barrier, 2)
    for kh in range(2):
        for r in range(2):
            pl.when(has_x1[r])(x1_copy(kh, r).start)

    ld_k[0].wait()
    for g in G:
        proj(x0[0], WK, 0, 0, g)
    ld_q[0].wait()
    for g in G:
        proj(x0[0], WQ, 0, 0, g)
    x1 = [x1_wait(0)]
    for w in (WK, WQ):
        for g in G:
            proj(x1[0], w, 1, 0, g)
    ld_k[1].wait()
    k0 = [proj(x0[1], WK, 0, 1, g).astype(BF) for g in G]
    x1.append(x1_wait(1))
    k1 = [proj(x1[1], WK, 1, 1, g).astype(BF) for g in G]
    ld_q[1].wait()
    q0 = [interleave_halves(proj(x0[1], WQ, 0, 1, g) * QSCALE) for g in G]
    p0 = [probs(q0[g], k0[g]) for g in G]
    q1 = [interleave_halves(proj(x1[1], WQ, 1, 1, g) * QSCALE) for g in G]

    for kh in range(2):
        for r in range(2):
            pl.when(has_x1[r])(x1_copy(kh, r).wait_send)
    ld_v[0].wait()
    r0 = [inv_sum(p0[g]) for g in G]
    for g in (0, 1):
        proj(x0[0], WV, 0, 0, g)
    p1 = [probs(q1[g], k1[g]) for g in G]
    for b, g in ((0, 2), (0, 3), (1, 0), (1, 1), (1, 2), (1, 3)):
        proj((x0, x1)[b][0], WV, b, 0, g)
    ld_v[1].wait()
    r1 = [inv_sum(p1[g]) for g in G]
    v0 = [proj(x0[1], WV, 0, 1, g).astype(BF) for g in G]
    v1 = [proj(x1[1], WV, 1, 1, 0, row_tiles=2).astype(BF)]
    o0 = [attend(p0[g], v0[g], r0[g]) for g in (0, 1)]
    o0 += [jnp.concatenate([attend(p0[g], v0[g], r0[g], t) for t in TILES], axis=0) for g in (2, 3)]
    o0 = jnp.concatenate(o0, axis=1)

    o_wait(0)
    pub = out_proj(o0, 0, 0)
    v1 += [proj(x1[1], WV, 1, 1, g).astype(BF) for g in (1, 2)]
    pub[0]()
    v1.append(proj(x1[1], WV, 1, 1, 3, row_tiles=2).astype(BF))
    run(*pub[1:])
    o_wait(1)
    pub = out_proj(o0, 0, 1)
    o1 = [jnp.concatenate([attend(p1[g], v1[g], r1[g], TILES[0]) for g in G], axis=1)]
    pub[0]()
    o1.append(jnp.concatenate([attend(p1[g], v1[g], r1[g], TILES[1]) for g in G], axis=1))
    run(*pub[1:])
    run(*[f for t in range(2) for c in (1, 0) for f in out_proj(o1[t], 1, c, t * UPH // 2)])
    o1 = jnp.concatenate(o1, axis=0)
    o_wait(2)
    run(*out_proj(o1, 1, 2), *out_proj(o0, 0, 2))
    o_wait(3)
    run(*out_proj(o0, 0, 3), *out_proj(o1, 1, 3))

    for uid, h, _, _ in own2:
        rcopy(0, uid, h).wait_recv()
        acc = part_v[uid] + rcv1[uid].astype(F32)
        snd2[uid] = acc.astype(BF)
        rcopy(1, uid, h).start()
        part_v[uid] = acc
    for n, (uid, h, row, col) in enumerate(own3):
        rcopy(0, *other[n][:2]).wait_send()
        rcopy(1, uid, h).wait()
        acc = part_v[uid] + rcv2[uid].astype(F32)
        snd3[uid] = acc.astype(BF)
        rcopy(2, uid, h).start()
        out_ref[pl.ds(row, UR), pl.ds(col, 128)] = acc
    for n, (uid, h, row, col) in enumerate(other):
        rcopy(2, *own3[n][:2]).wait_send()
        rcopy(2, uid, h).wait_recv()
        out_ref[pl.ds(row, UR), pl.ds(col, 128)] = rcv3[uid].astype(F32)


def pallas_dist_attn_self_mha_htp_b2_sq128_skv128_d512_hq8_dh64_kernel(x, Wq, Wk, Wv, Wo):
    unit_buf = pltpu.VMEM((NU, UR, 128), BF)
    out = pl.pallas_call(
        _body,
        out_shape=jax.ShapeDtypeStruct((M, D), F32),
        in_specs=[pl.BlockSpec(memory_space=pl.ANY)] * 5,
        out_specs=pl.BlockSpec(memory_space=pltpu.VMEM),
        scratch_shapes=[
            pltpu.VMEM((M, D), F32),
            pltpu.VMEM((2, 2, 2, HR, 128), BF),
            pltpu.VMEM((2, 256, D), F32),
            pltpu.VMEM((2, 256, D), F32),
            pltpu.VMEM((2, 256, D), F32),
            pltpu.VMEM((NC, 16, 32, 128), F32),
            pltpu.VMEM((3, B, NG, S, 128), F32),
            pltpu.VMEM((NU, UR, 128), F32),
            unit_buf, unit_buf, unit_buf, unit_buf, unit_buf, unit_buf,
            pltpu.SemaphoreType.DMA((9 + NC,)),
            pltpu.SemaphoreType.DMA((6,)),
            pltpu.SemaphoreType.DMA((NU,)),
            pltpu.SemaphoreType.DMA((2 * NU,)),
        ],
        compiler_params=pltpu.CompilerParams(collective_id=0, disable_semaphore_checks=True),
    )(x.reshape(M, D), Wq, Wk, Wv, Wo.reshape(16, 32, D))
    return out.reshape(B, S, D)
```
